```python
import numpy as np

kernel_name = "dist_sparse_attn_blocksparse_kvseq_b2_sq256_skv256_hq4_dh64"

def setup_inputs():
    x = np.random.randn(2, 256, 512).astype(np.float32)
    Wq = np.random.randn(512, 256).astype(np.float32) * 0.02
    K_ext = np.random.randn(2, 1024, 4, 64).astype(np.float32)
    V_ext = np.random.randn(2, 1024, 4, 64).astype(np.float32)
    Wo = np.random.randn(256, 512).astype(np.float32) * 0.02
    return {"x": x, "Wq": Wq, "K_ext": K_ext, "V_ext": V_ext, "Wo": Wo}

def reference(x, Wq, K_ext, V_ext, Wo):
    B, Sq, Skv, Hq, Dh = 2, 256, 1024, 4, 64
    Q = (x @ Wq).reshape(B, Sq, Hq, Dh)
    qb = (np.arange(Sq) // 64)[:, None]
    kb = (np.arange(Skv) // 64)[None, :]
    mask = (qb == kb) | (kb == 0) | ((qb + kb) % 3 == 0)
    scores = np.einsum('bihd,bjhd->bhij', Q, K_ext).astype(np.float32) * 0.125
    scores = np.where(mask[None, None, :, :], scores, -1e9)
    scores_max = scores.max(axis=-1, keepdims=True)
    w = np.exp(scores - scores_max)
    row_keep = mask.any(axis=1)
    w_sum = np.where(row_keep[None, None, :, None], w.sum(axis=-1, keepdims=True), 1.0)
    w = w / w_sum
    w = np.where(row_keep[None, None, :, None], w, 0.0)
    ctx = np.einsum('bhij,bjhd->bihd', w, V_ext).reshape(B, Sq, Hq * Dh)
    return ctx @ Wo
```

```python
import contextlib
import functools
import jax
import jax.numpy as jnp
from jax import lax
from jax.experimental import pallas as pl
from jax.experimental.pallas import tpu as pltpu

N_DEV = 4
B, SQ, DM, H, DH = 2, 256, 512, 4, 64
NEG = -1e9
LOG2E = 1.4426950408889634
f32 = jnp.float32
bf16 = jnp.bfloat16
MESH = pl.DeviceIdType.MESH
ALL = frozenset(range(4))
GROUP_QB = {0: (0, 3), 1: (1, 2)}
NT = (((1,), (1,)), ((), ()))
add = lambda xs: functools.reduce(lambda u, v: u + v, xs)


def _allowed(qb, kb):
    return qb == kb or kb == 0 or (qb + kb) % 3 == 0


def _key_blocks(chip, g):
    out = []
    for j in range(4):
        kb = 4 * chip + j
        a = tuple(_allowed(qb, kb) for qb in GROUP_QB[g])
        if any(a):
            out.append((j, a))
    return out


PIECES = [(b, g, p) for b in range(2) for g in range(2) for p in range(2)]
PID = {pc: i for i, pc in enumerate(PIECES)}


def path(a, b, c, d, fa=1, fd=1):
    F = frozenset
    return [(a, b, F([a])), (d, c, F([d])), (b, c, F([a, b])), (c, b, F([c, d])),
            (b, a, ALL if fa else F([b, c, d])), (c, d, ALL if fd else F([a, b, c]))]


def make_kernel(scheme, fwd, loads_order, steps, scopes=False):
    msgs = [(pc, s, d, ct) for pc in PIECES for (s, d, ct) in scheme[pc]]
    MID = {m: i for i, m in enumerate(msgs)}

    def is_kv(m):
        return len(m[3]) == 1 and m[0] in fwd.get(m[1], ())

    def nblk(m):
        return len(_key_blocks(m[1], m[0][1]))

    rslot, cnt = {}, [0] * 4
    for m in msgs:
        if m[3] != ALL:
            rslot[m] = cnt[m[2]]
            cnt[m[2]] += 2 * (nblk(m) if is_kv(m) else 1)
    nrs = max(cnt)
    sslot, cnt = {}, [0] * 4
    for m in msgs:
        pc, s, d, ct = m
        if ct != ALL and (pc, s, ct) not in sslot:
            sslot[(pc, s, ct)] = cnt[s]
            cnt[s] += 2 * (nblk(m) if is_kv(m) else 1)
    nss = max(cnt)
    NM = len(msgs)

    def kernel(x, Wq, K_ext, V_ext, Wo):
        kt = jnp.transpose(K_ext, (0, 2, 3, 1)).reshape(B * H * DH, SQ)
        vt = jnp.transpose(V_ext, (0, 2, 3, 1)).reshape(B * H * DH, SQ)
        x2 = x.reshape(B * SQ, DM)

        def body(x_hbm, wq_hbm, kt_hbm, vt_hbm, wo_hbm, out_ref,
                 xb, wqb, ktb, vtb, wob, sbuf, sstat, rbuf, rstat, fin,
                 lsem, s_sem, r_sem, rdy):
            my = lax.axis_index("i")
            bar = pltpu.get_barrier_semaphore()

            def program(c):
                nsc = [0]

                def scope(name):
                    nsc[0] += 1
                    return jax.named_scope(f"s{nsc[0]:02d}_{name}") if scopes else contextlib.nullcontext()

                loads = {}

                def ld(key, src, dst):
                    cp = pltpu.make_async_copy(src, dst, lsem.at[len(loads)])
                    cp.start()
                    loads[key] = [cp, False]

                alias = {}
                for ck in loads_order[c]:
                    kind = ck[0]
                    if kind == "w":
                        if len(ck) == 1:
                            ld(ck, wq_hbm, wqb)
                            alias[("w", 0)] = alias[("w", 1)] = [ck]
                        else:
                            sl = pl.ds(ck[1] * 128, 128)
                            ld(ck, wq_hbm.at[:, sl], wqb.at[:, sl])
                            alias[ck] = [ck]
                    elif kind == "x":
                        _, b, g = ck
                        if g == 0:
                            ld(ck + (0,), x_hbm.at[pl.ds(b * 256, 64)], xb.at[b * 2, pl.ds(0, 64)])
                            ld(ck + (1,), x_hbm.at[pl.ds(b * 256 + 192, 64)], xb.at[b * 2, pl.ds(64, 64)])
                            alias[ck] = [ck + (0,), ck + (1,)]
                        else:
                            ld(ck, x_hbm.at[pl.ds(b * 256 + 64, 128)], xb.at[b * 2 + 1])
                            alias[ck] = [ck]
                    elif kind in ("k", "v"):
                        _, bs, ps, ts = ck
                        src, dst = (kt_hbm, ktb) if kind == "k" else (vt_hbm, vtb)
                        r0 = bs[0] * 256 + ps[0] * 128
                        nr = (256 * len(bs)) if len(ps) == 2 else 128
                        assert len(ps) == 2 or len(bs) == 1
                        rows = pl.ds(r0, nr)
                        if len(ts) == 2:
                            ld(ck, src.at[rows], dst.at[rows])
                        else:
                            cols = pl.ds(ts[0] * 128, 128)
                            ld(ck, src.at[rows, cols], dst.at[rows, cols])
                        for b in bs:
                            for p in ps:
                                for t in ts:
                                    alias[(kind, b, p, t)] = [ck]
                    elif kind == "o":
                        ld(ck, wo_hbm, wob)
                        alias[ck] = [ck]

                known = set()
                if c == 0:
                    for d in (1, 3):
                        pl.semaphore_signal(bar, inc=1, device_id=(d,), device_id_type=MESH)
                elif c in (1, 3):
                    pl.semaphore_wait(bar, 1)
                    known.add(0)
                    pl.semaphore_signal(bar, inc=1, device_id=(2,), device_id_type=MESH)
                    pl.semaphore_signal(rdy.at[c], inc=1, device_id=(0,), device_id_type=MESH)
                else:
                    pl.semaphore_wait(bar, 2)
                    known.update((0, 1, 3))
                    for d in (1, 3, 0):
                        pl.semaphore_signal(rdy.at[2], inc=1, device_id=(d,), device_id_type=MESH)

                def know(d):
                    if d in known:
                        return
                    if c in (1, 3) and d in (1, 3):
                        d = 2
                    pl.semaphore_wait(rdy.at[d], 1)
                    known.add(d)
                    if d == 2:
                        known.update((1, 3) if c != 0 else ())

                def need(*keys):
                    todo = []
                    for key in keys:
                        for k in alias[key]:
                            if not loads[k][1]:
                                loads[k][1] = True
                                todo.append(k)
                    if todo:
                        with scope("L" + "".join(map(str, todo[-1])).replace(" ", "").replace(",", "").replace("(", "").replace(")", "")):
                            for k in todo:
                                loads[k][0].wait()

                lane64 = lax.broadcasted_iota(jnp.int32, (64, 128), 1) < 64
                lane128 = lax.broadcasted_iota(jnp.int32, (128, 128), 1) < 64
                lane256 = (lax.broadcasted_iota(jnp.int32, (64, 256), 1) % 128) < 64
                C = {}
                have = {pc + (h,): {} for pc in PIECES for h in range(2)}
                final = set()
                sent = set()
                started = []
                queue = []

                def rc(src, dst, k, d):
                    return pltpu.make_async_remote_copy(src, dst, s_sem.at[k], r_sem.at[k], device_id=(d,), device_id_type=MESH)

                def descs(m, h):
                    pc, s, d, ct = m
                    k = MID[m] * 4 + h * 2
                    if ct == ALL:
                        r = fin.at[PID[pc], pl.ds(h * 64, 64)]
                        return [rc(r, r, k, d)]
                    ss, rs = sslot[(pc, s, ct)], rslot[m]
                    if is_kv(m):
                        n = nblk(m)
                        return [rc(sbuf.at[pl.ds((ss + h * n) * 64, n * 64)], rbuf.at[pl.ds((rs + h * n) * 64, n * 64)], k, d)]
                    return [rc(sstat.at[ss + h], rstat.at[rs + h], k + 1, d),
                            rc(sbuf.at[pl.ds((ss + h) * 64, 64)], rbuf.at[pl.ds((rs + h) * 64, 64)], k, d)]

                def tag(m, h):
                    return "".join(map(str, m[0])) + f"h{h}_" + ("F" if m[3] == ALL else "".join(map(str, sorted(m[3]))))

                def go():
                    if not queue:
                        return
                    for m, h in queue:
                        know(m[2])
                    with scope("S" + "+".join(tag(m, h) + f">{m[2]}" for m, h in queue)):
                        for m, h in queue:
                            for dsc in descs(m, h):
                                dsc.start()
                                started.append(dsc)
                    queue.clear()

                def merge(parts):
                    m = functools.reduce(jnp.maximum, [pt[1] for pt in parts])
                    a = [jnp.exp2(pt[1] - m) for pt in parts]
                    l = add([ai * pt[2] for ai, pt in zip(a, parts)])
                    return m, a, l

                def get(key, ct):
                    hv = have[key]
                    rem, parts = set(ct), []
                    for k in sorted(hv, key=lambda k: -len(k)):
                        if k <= rem:
                            parts.append(hv[k])
                            rem -= k
                    return parts if not rem else None

                def flush(pc, do_final=True):
                    outs = [m for m in msgs if m[0] == pc and m[1] == c]
                    recv_final = any(m[0] == pc and m[2] == c and m[3] == ALL for m in msgs)
                    for h in range(2):
                        key = pc + (h,)
                        for m in outs:
                            ct = m[3]
                            if ct == ALL or is_kv(m) or (m, h) in sent:
                                continue
                            parts = get(key, ct)
                            if parts is None:
                                continue
                            if ("stored", key, ct) not in C:
                                if len(parts) > 1:
                                    mm, a, l = merge(parts)
                                    have[key][ct] = (add([ai * pt[0] for ai, pt in zip(a, parts)]), mm, l)
                                o, mm, l = have[key][ct]
                                ss = sslot[(pc, c, ct)] + h
                                sbuf[pl.ds(ss * 64, 64)] = o.astype(bf16)
                                sstat[ss, 0:1] = mm
                                sstat[ss, 1:2] = l
                                C[("stored", key, ct)] = True
                            sent.add((m, h))
                            queue.append((m, h))
                    if do_final and pc not in final and not recv_final:
                        pp = [get(pc + (h,), ALL) for h in range(2)]
                        if all(x is not None for x in pp):
                            o = []
                            for parts in pp:
                                mm, a, l = merge(parts)
                                inv = 1.0 / l
                                o.append(add([(ai * inv) * pt[0] for ai, pt in zip(a, parts)]))
                            t = jnp.concatenate(o, axis=0).T
                            if pc[1] == 1:
                                t = jnp.concatenate([jnp.where(lane64, t[0:64], t[64:128]),
                                                     jnp.where(lane64, t[64:128], t[0:64])], axis=0)
                            fin[PID[pc]] = t.astype(bf16)
                            final.add(pc)
                    if pc in final:
                        for m in outs:
                            for h in range(2):
                                if m[3] == ALL and (m, h) not in sent:
                                    sent.add((m, h))
                                    queue.append((m, h))

                def wait_msgs(lst):
                    lst = [(m, h) for m, h in lst if ("got", m, h) not in C]
                    if not lst:
                        return
                    with scope("R" + "+".join(tag(m, h) + f"<{m[1]}" for m, h in lst)):
                        for m, h in lst:
                            for dsc in descs(m, h):
                                dsc.wait_recv()
                            C[("got", m, h)] = True

                def g_of(step):
                    return step[2]

                def qb_keys(u):
                    return [j for j, a in _key_blocks(c, 1) if a[u]]

                def kv_in(pc):
                    return [m for m in msgs if m[0] == pc and m[2] == c and is_kv(m)]

                for step in steps[c]:
                    op = step[0]
                    if op == "need":
                        need(*step[1:])
                    elif op == "kprep":
                        need(*[("k", b, p, t) for b, p, ts in step[1] for t in ts])
                        for b, p, ts in step[1]:
                            kk = ktb[pl.ds(b * 256 + p * 128, 128), pl.ds(ts[0] * 128, 128 * len(ts))].T
                            for n_, t in enumerate(ts):
                                for jj in range(2):
                                    C[("k", b, p, 2 * t + jj)] = kk[n_ * 128 + jj * 64: n_ * 128 + jj * 64 + 64]
                    elif op == "kvK" or op == "kvV":
                        js = [j for j, _ in _key_blocks(c, 0)]
                        n = len(js)
                        if op == "kvV":
                            need(*[("v", b, p, j // 2) for b, p in step[1] for j in js])
                        for b, p in step[1]:
                            pc = (b, 0, p)
                            ss = sslot[(pc, c, frozenset([c]))]
                            if op == "kvK":
                                for n_, j in enumerate(js):
                                    sbuf[pl.ds((ss + n_) * 64, 64)] = C[("k", b, p, j)].astype(bf16)
                            elif n == 1:
                                j = js[0]
                                v = vtb[pl.ds(b * 256 + p * 128, 128), pl.ds((j // 2) * 128, 128)]
                                v0, v1 = v[0:64], v[64:128]
                                if j % 2 == 1:
                                    v0 = pltpu.roll(v0, 64, 1)
                                else:
                                    v1 = pltpu.roll(v1, 64, 1)
                                sbuf[pl.ds((ss + 1) * 64, 64)] = jnp.where(lane64, v0, v1).astype(bf16)
                            else:
                                assert js == [0, 3]
                                rows = pl.ds(b * 256 + p * 128, 128)
                                sbuf[pl.ds((ss + 2) * 64, 128)] = jnp.where(
                                    lane128, vtb[rows, 0:128], vtb[rows, 128:256]).astype(bf16)
                            for m in msgs:
                                if m[0] == pc and m[1] == c and is_kv(m):
                                    hh = 0 if op == "kvK" else 1
                                    sent.add((m, hh))
                                    queue.append((m, hh))
                    elif op == "wq":
                        ps = step[1]
                        need(*[("w", p) for p in ps])
                        for p in ps:
                            C[("w", p)] = wqb[:, pl.ds(p * 128, 128)].astype(bf16)
                    elif op == "xc":
                        _, b, g = step
                        need(("x", b, g))
                        C[("x", b, g)] = xb[b * 2 + g].astype(bf16)
                    elif op == "q":
                        _, b, g, ps = step
                        if ("x", b, g) not in C:
                            need(("x", b, g))
                            C[("x", b, g)] = xb[b * 2 + g].astype(bf16)
                        for p in ps:
                            qp = jnp.dot(C[("x", b, g)], C[("w", p)], preferred_element_type=f32) * (0.125 * LOG2E)
                            q0, q1 = jnp.where(lane128, qp, 0.0), jnp.where(lane128, 0.0, qp)
                            if g == 0:
                                tiles = [q0, q1]
                            elif c == 0:
                                tiles = [q0, q1[64:128], q1[0:64]]
                            else:
                                tiles = None
                                C[("q", b, g, p)] = [jnp.concatenate([q0[0:64], q1[0:64]], axis=0).astype(bf16),
                                                     jnp.concatenate([q1[64:128], q0[64:128]], axis=0).astype(bf16)]
                            if tiles is not None:
                                C[("q", b, g, p)] = jnp.concatenate(tiles, axis=0).astype(bf16)
                    elif op == "s" and g_of(step) == 1 and c != 0:
                        _, b, g, ps = step[:4]
                        split = step[4] if len(step) > 4 else 1
                        kbs = _key_blocks(c, g)
                        ss_ = {}
                        for p in ps:
                            for u in range(2):
                                js = qb_keys(u)
                                if split > 1:
                                    ss_[(p, u)] = jnp.concatenate([
                                        lax.dot_general(C[("k", b, p, j)].astype(bf16), C[("q", b, g, p)][u], NT,
                                                        preferred_element_type=f32) for j in js], axis=0)
                                else:
                                    kall = jnp.concatenate([C[("k", b, p, j)] for j in js], axis=0).astype(bf16)
                                    ss_[(p, u)] = lax.dot_general(kall, C[("q", b, g, p)][u], NT, preferred_element_type=f32)
                        for p in ps:
                            res = []
                            for u in range(2):
                                s = ss_[(p, u)]
                                m_ = jnp.max(s, axis=0, keepdims=True)
                                pt = jnp.exp2(s - m_)
                                res.append((pt, m_, jnp.sum(pt, axis=0, keepdims=True)))
                            C[("p", b, g, p)] = res
                    elif op == "pv" and g_of(step) == 1 and c != 0:
                        _, b, g, ps = step[:4]
                        split = step[4] if len(step) > 4 else 1
                        need(*[("v", b, p, t) for p in ps for t in range(2)])
                        zero = jnp.zeros((64, 128), f32)
                        for p in ps:
                            res = C[("p", b, g, p)]
                            rows = pl.ds(b * 256 + p * 128, 128)
                            oo = []
                            for u in range(2):
                                js = qb_keys(u)
                                pt = res[u][0]
                                if len(js) == 2:
                                    assert js == [0, 3]
                                    vv = jnp.where(lane128, vtb[rows, 0:128], vtb[rows, 128:256])
                                else:
                                    j = js[0]
                                    vv = vtb[rows, pl.ds((j // 2) * 128, 128)]
                                    pt = jnp.concatenate([pt, zero] if j % 2 == 0 else [zero, pt], axis=0)
                                ptb = pt.astype(bf16)
                                if split > 1:
                                    oo.append([jnp.dot(vv[h * 64:(h + 1) * 64].astype(bf16), ptb, preferred_element_type=f32)
                                               for h in range(2)])
                                else:
                                    o = jnp.dot(vv.astype(bf16), ptb, preferred_element_type=f32)
                                    oo.append([o[0:64], o[64:128]])
                            l1 = lane64[0:1]
                            for h in range(2):
                                a_, b_ = (0, 1) if h == 0 else (1, 0)
                                have[(b, g, p, h)][frozenset([c])] = (
                                    jnp.where(lane64, oo[a_][h], oo[b_][h]),
                                    jnp.where(l1, res[a_][1], res[b_][1]), jnp.where(l1, res[a_][2], res[b_][2]))
                    elif op == "s":
                        _, b, g, ps = step[:4]
                        split = step[4] if len(step) > 4 else 1
                        kbs = _key_blocks(c, g)
                        wait_msgs([(m, 0) for p in ps for m in kv_in((b, g, p))])
                        ss_ = {}
                        for p in ps:
                            pc = (b, g, p)
                            qm = C[("q", b, g, p)]
                            kall = jnp.concatenate([C[("k", b, p, j)] for j, _ in kbs], axis=0)
                            nk = kall.shape[0] // split
                            s = jnp.concatenate([
                                lax.dot_general(kall[i * nk:(i + 1) * nk].astype(bf16), qm, NT, preferred_element_type=f32)
                                for i in range(split)], axis=0)
                            blocks = []
                            for n_, (j, a) in enumerate(kbs):
                                sb = s[n_ * 64:(n_ + 1) * 64]
                                if not a[0]:
                                    sb = jnp.where(lane256, NEG, sb)
                                if not a[1]:
                                    sb = jnp.where(lane256, sb, NEG)
                                blocks.append(sb)
                            for m in kv_in(pc):
                                blocks.append(lax.dot_general(rbuf[pl.ds(rslot[m] * 64, nblk(m) * 64)], qm, NT,
                                                              preferred_element_type=f32))
                            ss_[p] = blocks
                        for p in ps:
                            s = jnp.concatenate(ss_[p], axis=0)
                            m_ = jnp.max(s, axis=0, keepdims=True)
                            pt = jnp.exp2(s - m_)
                            l = jnp.sum(pt, axis=0, keepdims=True)
                            C[("p", b, g, p)] = (pt, m_, l)
                    elif op == "pv":
                        _, b, g, ps = step[:4]
                        js = [j for j, _ in _key_blocks(c, g)]
                        need(*[("v", b, p, j // 2) for p in ps for j in js])
                        wait_msgs([(m, 1) for p in ps for m in kv_in((b, g, p))])
                        zero = jnp.zeros((64, 128), f32)
                        for p in ps:
                            pc = (b, g, p)
                            pt, m_, l = C[("p", b, g, p)]
                            for h in range(2):
                                r0 = b * 256 + p * 128 + h * 64
                                cols = slice(h * 128, (h + 1) * 128)
                                rows = {j: pt[n_ * 64:(n_ + 1) * 64, cols] for n_, j in enumerate(js)}
                                terms = []
                                if set(js) in ({0, 3}, {1, 2}):
                                    ev = [j for j in js if j % 2 == 0][0]
                                    od = [j for j in js if j % 2 == 1][0]
                                    vsel = jnp.where(lane64, vtb[pl.ds(r0, 64), pl.ds((ev // 2) * 128, 128)],
                                                     vtb[pl.ds(r0, 64), pl.ds((od // 2) * 128, 128)])
                                    terms.append((vsel.astype(bf16), jnp.concatenate([rows[ev], rows[od]], axis=0)))
                                else:
                                    for t in range(2):
                                        if 2 * t in rows or 2 * t + 1 in rows:
                                            terms.append((vtb[pl.ds(r0, 64), pl.ds(t * 128, 128)].astype(bf16),
                                                          jnp.concatenate([rows.get(2 * t, zero), rows.get(2 * t + 1, zero)], axis=0)))
                                off = len(js) * 64
                                for m in kv_in(pc):
                                    n = nblk(m)
                                    pr = pt[off:off + n * 64, cols]
                                    off += n * 64
                                    if n == 1:
                                        terms.append((rbuf[pl.ds((rslot[m] + 1) * 64, 64)],
                                                      jnp.concatenate([pr, zero] if h == 0 else [zero, pr], axis=0)))
                                    else:
                                        terms.append((rbuf[pl.ds((rslot[m] + 2 + h) * 64, 64)], pr))
                                o = add([jnp.dot(vv, pp.astype(bf16), preferred_element_type=f32) for vv, pp in terms])
                                ct = frozenset([c] + [m[1] for m in kv_in(pc)])
                                have[pc + (h,)][ct] = (o, m_[:, cols], l[:, cols])
                    elif op == "recv":
                        lst = []
                        for b, g, p, src, hs in step[1]:
                            pc = (b, g, p)
                            for h in hs:
                                m = [m for m in msgs if m[0] == pc and m[1] == src and m[2] == c and not is_kv(m)
                                     and ("got", m, h) not in C][0]
                                lst.append((m, h))
                        wait_msgs(lst)
                        for m, h in lst:
                            if m[3] == ALL:
                                if all(("got", m, k) in C for k in range(2)):
                                    final.add(m[0])
                            else:
                                rs = rslot[m] + h
                                have[m[0] + (h,)][m[3]] = (rbuf[pl.ds(rs * 64, 64)].astype(f32), rstat[rs, 0:1], rstat[rs, 1:2])
                    elif op == "flush":
                        for pc in step[1]:
                            flush(pc)
                        go()
                    elif op == "stage":
                        for pc in step[1]:
                            flush(pc)
                    elif op == "fwd":
                        for pc in step[1]:
                            flush(pc, do_final=False)
                        go()
                    elif op == "go":
                        go()
                    elif op == "drain":
                        n = len(started) - step[1]
                        for dsc in started[:n]:
                            dsc.wait_send()
                        del started[:n]
                    elif op == "wo":
                        need(("o",))
                        C["wo"] = [wob[0:128, :].astype(bf16), wob[128:256, :].astype(bf16)]
                    elif op == "out":
                        _, b, g, ps = step
                        assert all((b, g, p) in final for p in ps), (c, step)
                        terms = [jnp.dot(fin[PID[(b, g, p)]], C["wo"][p], preferred_element_type=f32) for p in ps]
                        if ("acc", b, g) in C:
                            terms.append(C.pop(("acc", b, g)))
                        elif len(ps) == 1:
                            C[("acc", b, g)] = terms[0]
                            continue
                        o = add(terms)
                        if g == 0:
                            out_ref[b, 0:64, :] = o[0:64]
                            out_ref[b, 192:256, :] = o[64:128]
                        else:
                            out_ref[b, 64:192, :] = o
                        C[("done", b, g)] = True
                    else:
                        raise ValueError(step)
                assert not queue
                miss = [(m, h) for m in msgs for h in range(2) if m[1] == c and (m, h) not in sent]
                assert not miss, (c, miss)
                miss = [(m, h) for m in msgs for h in range(2) if m[2] == c and ("got", m, h) not in C]
                assert not miss, (c, miss)
                assert all(v[1] for v in loads.values()), (c, [k for k, v in loads.items() if not v[1]])
                assert all(("done", b, g) in C for b in range(2) for g in range(2)), c
                for d in ((1, 2, 3) if c == 0 else (2,) if c != 2 else ()):
                    know(d)
                with scope("end"):
                    for dsc in started:
                        dsc.wait_send()

            for c in range(N_DEV):
                pl.when(my == c)(functools.partial(program, c))

        return pl.pallas_call(
            body,
            out_shape=jax.ShapeDtypeStruct((B, SQ, DM), f32),
            in_specs=[pl.BlockSpec(memory_space=pl.ANY)] * 5,
            out_specs=pl.BlockSpec(memory_space=pltpu.VMEM),
            scratch_shapes=[
                pltpu.VMEM((4, 128, DM), f32), pltpu.VMEM((DM, 256), f32),
                pltpu.VMEM((512, 256), f32), pltpu.VMEM((512, 256), f32), pltpu.VMEM((256, DM), f32),
                pltpu.VMEM((nss * 64, 128), bf16), pltpu.VMEM((nss, 2, 128), f32),
                pltpu.VMEM((nrs * 64, 128), bf16), pltpu.VMEM((nrs, 2, 128), f32),
                pltpu.VMEM((8, 128, 128), bf16),
                pltpu.SemaphoreType.DMA((32,)),
                pltpu.SemaphoreType.DMA((NM * 4,)), pltpu.SemaphoreType.DMA((NM * 4,)),
                pltpu.SemaphoreType.REGULAR((4,)),
            ],
            compiler_params=pltpu.CompilerParams(collective_id=0, disable_bounds_checks=True,
                                                 disable_semaphore_checks=True),
        )(x2, Wq, kt, vt, Wo)

    return kernel


P01 = (0, 1)
H01 = (0, 1)
def plan():
    scheme = {}
    for p in range(2):
        scheme[(0,0,p)] = path(3,0,1,2)
        scheme[(1,0,p)] = path(2,3,0,1)
        scheme[(0,1,p)] = path(0,1,2,3,fa=0,fd=1)
        scheme[(1,1,p)] = path(1,2,3,0,fa=1,fd=0)
    fwd = {2: {(b,0,p) for b in range(2) for p in range(2)}, 1: {(1,0,0),(1,0,1)}, 3: {(0,0,0),(0,0,1)}}
    loads = {}; steps = {}
    for c, f in ((1, 1), (3, 0)):
        s = 1 - f
        loads[c] = [("k",(f,),(0,),P01), ("v",(f,),(0,),P01), ("w",0), ("x",f,1), ("k",(f,),(1,),P01), ("v",(f,),(1,),P01), ("w",1),
                    ("k",(s,),P01,P01), ("x",s,0), ("x",s,1), ("v",(s,),P01,P01), ("o",)]
        steps[c] = [("kprep",[(f,0,P01)]), ("kvK",[(f,0)]), ("kvV",[(f,0)]), ("go",),
                    ("wq",(0,)), ("q",f,1,(0,)),
                    ("kprep",[(f,1,P01)]), ("s",f,1,(0,),2), ("kvK",[(f,1)]), ("kvV",[(f,1)]), ("pv",f,1,(0,)), ("flush",[(f,1,0)]),
                    ("wq",(1,)), ("q",f,1,(1,)), ("kprep",[(s,0,P01),(s,1,P01)]), ("s",f,1,(1,),2), ("pv",f,1,(1,)), ("flush",[(f,1,1)]),
                    ("q",s,0,P01), ("xc",s,1), ("s",s,0,P01), ("q",s,1,P01), ("pv",s,0,P01), ("s",s,1,P01), ("flush",[(s,0,0),(s,0,1)]),
                    ("recv",[(s,1,0,0,H01),(s,1,1,0,H01)]), ("pv",s,1,P01), ("flush",[(s,1,0),(s,1,1)]),
                    ("wo",),
                    ("recv",[(s,1,0,2,(0,))]), ("fwd",[(s,1,0)]), ("recv",[(s,1,0,2,(1,))]), ("fwd",[(s,1,0)]),
                    ("recv",[(s,1,1,2,(0,))]), ("fwd",[(s,1,1)]), ("recv",[(s,1,1,2,(1,))]), ("fwd",[(s,1,1)]),
                    ("recv",[(s,0,0,0,H01),(s,0,1,0,H01)]), ("flush",[(s,0,0),(s,0,1),(s,1,0),(s,1,1)]),
                    ("out",s,0,P01), ("out",s,1,P01),
                    ("recv",[(f,0,0,0,H01),(f,0,1,0,H01)]), ("out",f,0,P01),
                    ("recv",[(f,1,0,2,H01),(f,1,1,2,H01)]), ("out",f,1,P01)]
    loads[0] = [("k",(0,),P01,P01), ("w",), ("x",0,1), ("v",(0,),P01,P01), ("k",(1,),P01,P01), ("x",1,1), ("v",(1,),P01,P01), ("x",1,0), ("x",0,0), ("o",)]
    steps[0] = [("kprep",[(0,0,P01),(0,1,P01)]), ("wq",P01), ("q",0,1,P01), ("s",0,1,P01),
                ("kprep",[(1,0,P01),(1,1,P01)]), ("pv",0,1,P01), ("flush",[(0,1,0),(0,1,1)]),
                ("q",1,1,P01), ("s",1,1,P01), ("xc",1,0), ("pv",1,1,P01), ("q",1,0,P01), ("flush",[(1,1,0),(1,1,1)]),
                ("q",0,0,P01), ("wo",),
                ("s",1,0,(0,),2), ("pv",1,0,(0,)), ("flush",[(1,0,0)]),
                ("s",0,0,(0,),2), ("pv",0,0,(0,)), ("flush",[(0,0,0)]),
                ("s",1,0,(1,),2), ("pv",1,0,(1,)), ("flush",[(1,0,1)]),
                ("s",0,0,(1,),2), ("pv",0,0,(1,)), ("flush",[(0,0,1)]),
                ("recv",[(0,0,0,1,H01),(1,0,0,3,H01)]), ("flush",[(0,0,0),(1,0,0)]),
                ("recv",[(0,0,1,1,H01),(1,0,1,3,H01)]), ("flush",[(0,0,1),(1,0,1)]),
                ("out",0,0,P01), ("out",1,0,P01),
                ("recv",[(0,1,0,1,H01),(1,1,0,3,H01)]), ("flush",[(0,1,0),(1,1,0)]), ("out",0,1,(0,)), ("out",1,1,(0,)),
                ("recv",[(0,1,1,1,H01),(1,1,1,3,H01)]), ("flush",[(0,1,1),(1,1,1)]), ("out",0,1,(1,)), ("out",1,1,(1,))]
    BP = [(0,0),(1,0),(0,1),(1,1)]
    loads[2] = [("k",(0,1),P01,(0,)), ("v",(0,1),P01,(0,)), ("w",0), ("x",0,1), ("k",(0,1),P01,(1,)), ("x",1,1), ("w",1), ("v",(0,1),P01,(1,)), ("o",)]
    steps[2] = [("kprep",[(b,p,(0,)) for b,p in BP]), ("kvK",[(0,0),(1,0)]), ("go",),
                ("kvV",[(0,0),(1,0)]), ("kvK",[(0,1),(1,1)]), ("kvV",[(0,1),(1,1)]), ("go",),
                ("wq",(0,)), ("q",0,1,(0,)), ("kprep",[(b,p,(1,)) for b,p in BP]), ("xc",1,1), ("s",0,1,(0,),2), ("q",1,1,(0,)),
                ("wq",(1,)), ("s",1,1,(0,),2), ("q",0,1,(1,)), ("q",1,1,(1,)),
                ("pv",0,1,(0,)), ("pv",1,1,(0,)), ("s",0,1,(1,)), ("s",1,1,(1,)),
                ("recv",[(0,1,0,3,H01),(1,1,0,1,H01)]), ("fwd",[(0,1,0),(1,1,0)]),
                ("pv",0,1,(1,)), ("pv",1,1,(1,)),
                ("recv",[(0,1,1,3,H01),(1,1,1,1,H01)]), ("fwd",[(0,1,1),(1,1,1)]),
                ("wo",),
                ("recv",[(0,1,0,1,H01),(1,1,0,3,H01)]), ("flush",[(0,1,0),(1,1,0)]),
                ("recv",[(0,1,1,1,H01),(1,1,1,3,H01)]), ("flush",[(0,1,1),(1,1,1)]),
                ("out",0,1,P01), ("out",1,1,P01),
                ("recv",[(0,0,0,1,H01),(0,0,1,1,H01)]), ("out",0,0,P01),
                ("recv",[(1,0,0,3,H01),(1,0,1,3,H01)]), ("out",1,0,P01)]
    return scheme, fwd, loads, steps


def pallas_dist_sparse_attn_blocksparse_kvseq_b2_sq256_skv256_hq4_dh64_kernel(x, Wq, K_ext, V_ext, Wo):
    return make_kernel(*plan())(x, Wq, K_ext, V_ext, Wo)
```

```python
import contextlib
import functools
import jax
import jax.numpy as jnp
from jax import lax
from jax.experimental import pallas as pl
from jax.experimental.pallas import tpu as pltpu

N_DEV = 4
B, SQ, DM, H, DH = 2, 256, 512, 4, 64
NEG = -1e9
LOG2E = 1.4426950408889634
f32 = jnp.float32
bf16 = jnp.bfloat16
MESH = pl.DeviceIdType.MESH
ALL = frozenset(range(4))
GROUP_QB = {0: (0, 3), 1: (1, 2)}
NT = (((1,), (1,)), ((), ()))
add = lambda xs: functools.reduce(lambda u, v: u + v, xs)


def _allowed(qb, kb):
    return qb == kb or kb == 0 or (qb + kb) % 3 == 0


def _key_blocks(chip, g):
    out = []
    for j in range(4):
        kb = 4 * chip + j
        a = tuple(_allowed(qb, kb) for qb in GROUP_QB[g])
        if any(a):
            out.append((j, a))
    return out


PIECES = [(b, g, p) for b in range(2) for g in range(2) for p in range(2)]
PID = {pc: i for i, pc in enumerate(PIECES)}


def path(a, b, c, d, fa=1, fd=1):
    F = frozenset
    return [(a, b, F([a])), (d, c, F([d])), (b, c, F([a, b])), (c, b, F([c, d])),
            (b, a, ALL if fa else F([b, c, d])), (c, d, ALL if fd else F([a, b, c]))]


def make_kernel(scheme, fwd, loads_order, steps, fine=(), scopes=False):
    msgs = [(pc, s, d, ct) for pc in PIECES for (s, d, ct) in scheme[pc]]
    MID = {m: i for i, m in enumerate(msgs)}

    def nsub(pc):
        return 4 if pc in fine else 2

    def nparts(m):
        return 2 if (m[3] == ALL or is_kv(m)) else nsub(m[0])

    def is_kv(m):
        return len(m[3]) == 1 and m[0] in fwd.get(m[1], ())

    def nblk(m):
        return len(_key_blocks(m[1], m[0][1]))

    rslot, cnt = {}, [0] * 4
    for m in msgs:
        if m[3] != ALL:
            rslot[m] = cnt[m[2]]
            cnt[m[2]] += 2 * (nblk(m) if is_kv(m) else 1)
    nrs = max(cnt)
    sslot, cnt = {}, [0] * 4
    for m in msgs:
        pc, s, d, ct = m
        if ct != ALL and (pc, s, ct) not in sslot:
            sslot[(pc, s, ct)] = cnt[s]
            cnt[s] += 2 * (nblk(m) if is_kv(m) else 1)
    nss = max(cnt)
    ssem_id, rsem_id = {}, {}
    sc, rc_ = [0] * 4, [0] * 4
    for m in msgs:
        for u in range(nparts(m)):
            for kind in range(2):
                if kind == 1 and (m[3] == ALL or is_kv(m) or (nparts(m) == 4 and u % 2 == 1)):
                    continue
                ssem_id[(m, u, kind)] = sc[m[1]]
                rsem_id[(m, u, kind)] = rc_[m[2]]
                sc[m[1]] += 1
                rc_[m[2]] += 1
    NSS, NRS = max(sc), max(rc_)

    def kernel(x, Wq, K_ext, V_ext, Wo):
        kt = jnp.transpose(K_ext, (0, 2, 3, 1)).reshape(B * H * DH, SQ)
        vt = jnp.transpose(V_ext, (0, 2, 3, 1)).reshape(B * H * DH, SQ)
        x2 = x.reshape(B * SQ, DM)

        def body(x_hbm, wq_hbm, kt_hbm, vt_hbm, wo_hbm, out_ref,
                 xb, wqb, ktb, vtb, wob, sbuf, sstat, rbuf, rstat, fin,
                 lsem, s_sem, r_sem, rdy):
            my = lax.axis_index("i")
            bar = pltpu.get_barrier_semaphore()

            def program(c):
                nsc = [0]

                def scope(name):
                    nsc[0] += 1
                    on = scopes and (scopes is True or name[0] in scopes)
                    return jax.named_scope(f"s{nsc[0]:02d}_{name}") if on else contextlib.nullcontext()

                loads = {}

                def ld(key, src, dst):
                    cp = pltpu.make_async_copy(src, dst, lsem.at[len(loads)])
                    cp.start()
                    loads[key] = [cp, False]

                alias = {}
                for ck in loads_order[c]:
                    kind = ck[0]
                    if kind == "w":
                        if len(ck) == 1:
                            ld(ck, wq_hbm, wqb)
                            alias[("w", 0)] = alias[("w", 1)] = [ck]
                        else:
                            sl = pl.ds(ck[1] * 128, 128)
                            ld(ck, wq_hbm.at[:, sl], wqb.at[:, sl])
                            alias[ck] = [ck]
                    elif kind == "x":
                        _, b, g = ck
                        if g == 0:
                            ld(ck + (0,), x_hbm.at[pl.ds(b * 256, 64)], xb.at[b * 2, pl.ds(0, 64)])
                            ld(ck + (1,), x_hbm.at[pl.ds(b * 256 + 192, 64)], xb.at[b * 2, pl.ds(64, 64)])
                            alias[ck] = [ck + (0,), ck + (1,)]
                        else:
                            ld(ck, x_hbm.at[pl.ds(b * 256 + 64, 128)], xb.at[b * 2 + 1])
                            alias[ck] = [ck]
                    elif kind in ("k", "v"):
                        _, bs, ps, ts = ck
                        src, dst = (kt_hbm, ktb) if kind == "k" else (vt_hbm, vtb)
                        r0 = bs[0] * 256 + ps[0] * 128
                        nr = (256 * len(bs)) if len(ps) == 2 else 128
                        assert len(ps) == 2 or len(bs) == 1
                        rows = pl.ds(r0, nr)
                        if len(ts) == 2:
                            ld(ck, src.at[rows], dst.at[rows])
                        else:
                            cols = pl.ds(ts[0] * 128, 128)
                            ld(ck, src.at[rows, cols], dst.at[rows, cols])
                        for b in bs:
                            for p in ps:
                                for t in ts:
                                    alias[(kind, b, p, t)] = [ck]
                    elif kind == "o":
                        ld(ck, wo_hbm, wob)
                        alias[ck] = [ck]

                known = set()
                if c == 0:
                    for d in (1, 3):
                        pl.semaphore_signal(bar, inc=1, device_id=(d,), device_id_type=MESH)
                elif c in (1, 3):
                    pl.semaphore_wait(bar, 1)
                    known.add(0)
                    pl.semaphore_signal(bar, inc=1, device_id=(2,), device_id_type=MESH)
                    pl.semaphore_signal(rdy.at[c], inc=1, device_id=(0,), device_id_type=MESH)
                else:
                    pl.semaphore_wait(bar, 2)
                    known.update((0, 1, 3))
                    for d in (1, 3, 0):
                        pl.semaphore_signal(rdy.at[2], inc=1, device_id=(d,), device_id_type=MESH)

                def know(d):
                    if d in known:
                        return
                    if c in (1, 3) and d in (1, 3):
                        d = 2
                    pl.semaphore_wait(rdy.at[d], 1)
                    known.add(d)
                    if d == 2:
                        known.update((1, 3) if c != 0 else ())

                def need(*keys):
                    order = list(loads)
                    last = max(order.index(k) for key in keys for k in alias[key])
                    todo = [k for k in order[:last + 1] if not loads[k][1]]
                    if todo:
                        with scope("L" + "".join(map(str, todo[-1])).replace(" ", "").replace(",", "").replace("(", "").replace(")", "")):
                            for k in todo:
                                loads[k][1] = True
                                loads[k][0].wait()

                lane64 = lax.broadcasted_iota(jnp.int32, (64, 128), 1) < 64
                lane128 = lax.broadcasted_iota(jnp.int32, (128, 128), 1) < 64
                lane256 = (lax.broadcasted_iota(jnp.int32, (64, 256), 1) % 128) < 64
                C = {}
                have = {pc + (u,): {} for pc in PIECES for u in range(nsub(pc))}
                final = set()
                sent = set()
                started = []
                queue = []

                def rc(src, dst, k, d):
                    return pltpu.make_async_remote_copy(src, dst, s_sem.at[ssem_id[k]], r_sem.at[rsem_id[k]],
                                                        device_id=(d,), device_id_type=MESH)

                def put(pc, h, ct, o, m_, l):
                    if nsub(pc) == 2:
                        have[pc + (h,)][ct] = (o, m_, l)
                    else:
                        for i in range(2):
                            have[pc + (2 * h + i,)][ct] = (o[32 * i:32 * i + 32], m_, l)

                def descs(m, h):
                    pc, s, d, ct = m
                    if ct == ALL:
                        r = fin.at[PID[pc], pl.ds(h * 64, 64)]
                        return [rc(r, r, (m, h, 0), d)]
                    ss, rs = sslot[(pc, s, ct)], rslot[m]
                    if is_kv(m):
                        n = nblk(m)
                        return [rc(sbuf.at[pl.ds((ss + h * n) * 64, n * 64)], rbuf.at[pl.ds((rs + h * n) * 64, n * 64)], (m, h, 0), d)]
                    nr = 128 // nsub(pc)
                    hd = h * nr // 64
                    out = []
                    if (m, h, 1) in ssem_id:
                        out.append(rc(sstat.at[ss + hd], rstat.at[rs + hd], (m, h, 1), d))
                    out.append(rc(sbuf.at[pl.ds(ss * 64 + h * nr, nr)], rbuf.at[pl.ds(rs * 64 + h * nr, nr)], (m, h, 0), d))
                    return out

                def tag(m, h):
                    return "".join(map(str, m[0])) + f"h{h}_" + ("F" if m[3] == ALL else "".join(map(str, sorted(m[3]))))

                def go():
                    if not queue:
                        return
                    for m, h in queue:
                        know(m[2])
                    with scope("S" + "+".join(tag(m, h) + f">{m[2]}" for m, h in queue)):
                        for m, h in queue:
                            for dsc in descs(m, h):
                                dsc.start()
                                started.append(dsc)
                    queue.clear()

                def merge(parts):
                    m = functools.reduce(jnp.maximum, [pt[1] for pt in parts])
                    a = [jnp.exp2(pt[1] - m) for pt in parts]
                    l = add([ai * pt[2] for ai, pt in zip(a, parts)])
                    return m, a, l

                def get(key, ct):
                    hv = have[key]
                    rem, parts = set(ct), []
                    for k in sorted(hv, key=lambda k: -len(k)):
                        if k <= rem:
                            parts.append(hv[k])
                            rem -= k
                    return parts if not rem else None

                def flush(pc, do_final=True, head=None):
                    outs = [m for m in msgs if m[0] == pc and m[1] == c]
                    recv_final = any(m[0] == pc and m[2] == c and m[3] == ALL for m in msgs)
                    nr = 128 // nsub(pc)
                    for h in range(nsub(pc)):
                        if head is not None and h * nr // 64 != head:
                            continue
                        key = pc + (h,)
                        for m in outs:
                            ct = m[3]
                            if ct == ALL or is_kv(m) or (m, h) in sent:
                                continue
                            parts = get(key, ct)
                            if parts is None:
                                continue
                            if ("stored", key, ct) not in C:
                                if len(parts) > 1:
                                    mm, a, l = merge(parts)
                                    have[key][ct] = (add([ai * pt[0] for ai, pt in zip(a, parts)]), mm, l)
                                o, mm, l = have[key][ct]
                                ss = sslot[(pc, c, ct)]
                                sbuf[pl.ds(ss * 64 + h * nr, nr)] = o.astype(bf16)
                                if (h * nr) % 64 == 0:
                                    sstat[ss + h * nr // 64, 0:1] = mm
                                    sstat[ss + h * nr // 64, 1:2] = l
                                C[("stored", key, ct)] = True
                            sent.add((m, h))
                            queue.append((m, h))
                    if do_final and pc not in final and not recv_final:
                        pp = [get(pc + (h,), ALL) for h in range(nsub(pc))]
                        if all(x is not None for x in pp):
                            o = []
                            for parts in pp:
                                mm, a, l = merge(parts)
                                inv = 1.0 / l
                                o.append(add([(ai * inv) * pt[0] for ai, pt in zip(a, parts)]))
                            t = jnp.concatenate(o, axis=0).T
                            fin[PID[pc]] = t.astype(bf16)
                            final.add(pc)
                    if pc in final:
                        for m in outs:
                            for h in range(2):
                                if m[3] == ALL and (m, h) not in sent:
                                    sent.add((m, h))
                                    queue.append((m, h))

                def wait_msgs(lst):
                    lst = [(m, h) for m, h in lst if ("got", m, h) not in C]
                    if not lst:
                        return
                    with scope("R" + "+".join(tag(m, h) + f"<{m[1]}" for m, h in lst)):
                        for m, h in lst:
                            for dsc in descs(m, h):
                                dsc.wait_recv()
                            C[("got", m, h)] = True

                def g_of(step):
                    return step[2]

                def qb_keys(u):
                    return [j for j, a in _key_blocks(c, 1) if a[u]]

                def kv_in(pc):
                    return [m for m in msgs if m[0] == pc and m[2] == c and is_kv(m)]

                for step in steps[c]:
                    op = step[0]
                    if op == "need":
                        need(*step[1:])
                    elif op == "kvw":
                        wait_msgs([(m, part) for b, p, part in step[1] for m in kv_in((b, 0, p))])
                    elif op == "kprep":
                        need(*[("k", b, p, t) for b, p, ts in step[1] for t in ts])
                        for b, p, ts in step[1]:
                            kk = ktb[pl.ds(b * 256 + p * 128, 128), pl.ds(ts[0] * 128, 128 * len(ts))].T
                            for n_, t in enumerate(ts):
                                for jj in range(2):
                                    C[("k", b, p, 2 * t + jj)] = kk[n_ * 128 + jj * 64: n_ * 128 + jj * 64 + 64]
                    elif op == "kvK" or op == "kvV":
                        js = [j for j, _ in _key_blocks(c, 0)]
                        n = len(js)
                        if op == "kvV":
                            need(*[("v", b, p, j // 2) for b, p in step[1] for j in js])
                        for b, p in step[1]:
                            pc = (b, 0, p)
                            ss = sslot[(pc, c, frozenset([c]))]
                            if op == "kvK":
                                for n_, j in enumerate(js):
                                    sbuf[pl.ds((ss + n_) * 64, 64)] = C[("k", b, p, j)].astype(bf16)
                            elif n == 1:
                                j = js[0]
                                v = vtb[pl.ds(b * 256 + p * 128, 128), pl.ds((j // 2) * 128, 128)]
                                v0, v1 = v[0:64], v[64:128]
                                if j % 2 == 1:
                                    v0 = pltpu.roll(v0, 64, 1)
                                else:
                                    v1 = pltpu.roll(v1, 64, 1)
                                sbuf[pl.ds((ss + 1) * 64, 64)] = jnp.where(lane64, v0, v1).astype(bf16)
                            else:
                                assert js == [0, 3]
                                rows = pl.ds(b * 256 + p * 128, 128)
                                sbuf[pl.ds((ss + 2) * 64, 128)] = jnp.where(
                                    lane128, vtb[rows, 0:128], vtb[rows, 128:256]).astype(bf16)
                            for m in msgs:
                                if m[0] == pc and m[1] == c and is_kv(m):
                                    hh = 0 if op == "kvK" else 1
                                    sent.add((m, hh))
                                    queue.append((m, hh))
                    elif op == "wq":
                        ps = step[1]
                        need(*[("w", p) for p in ps])
                        for p in ps:
                            C[("w", p)] = wqb[:, pl.ds(p * 128, 128)].astype(bf16)
                    elif op == "xc":
                        _, b, g = step
                        need(("x", b, g))
                        C[("x", b, g)] = xb[b * 2 + g].astype(bf16)
                    elif op == "q":
                        _, b, g, ps = step
                        if ("x", b, g) not in C:
                            need(("x", b, g))
                            C[("x", b, g)] = xb[b * 2 + g].astype(bf16)
                        for p in ps:
                            qp = jnp.dot(C[("x", b, g)], C[("w", p)], preferred_element_type=f32) * (0.125 * LOG2E)
                            q0, q1 = jnp.where(lane128, qp, 0.0), jnp.where(lane128, 0.0, qp)
                            if g == 0 or c == 0:
                                tiles = [q0, q1]
                            else:
                                tiles = None
                                C[("q", b, g, p)] = [jnp.concatenate([q0[0:64], q1[0:64]], axis=0).astype(bf16),
                                                     jnp.concatenate([q1[64:128], q0[64:128]], axis=0).astype(bf16)]
                            if tiles is not None:
                                C[("q", b, g, p)] = jnp.concatenate(tiles, axis=0).astype(bf16)
                    elif op == "s" and g_of(step) == 1 and c != 0:
                        _, b, g, ps = step[:4]
                        split = step[4] if len(step) > 4 else 1
                        kbs = _key_blocks(c, g)
                        ss_ = {}
                        for p in ps:
                            for u in range(2):
                                js = qb_keys(u)
                                if split > 1:
                                    ss_[(p, u)] = jnp.concatenate([
                                        lax.dot_general(C[("k", b, p, j)].astype(bf16), C[("q", b, g, p)][u], NT,
                                                        preferred_element_type=f32) for j in js], axis=0)
                                else:
                                    kall = jnp.concatenate([C[("k", b, p, j)] for j in js], axis=0).astype(bf16)
                                    ss_[(p, u)] = lax.dot_general(kall, C[("q", b, g, p)][u], NT, preferred_element_type=f32)
                        for p in ps:
                            res = []
                            for u in range(2):
                                s = ss_[(p, u)]
                                m_ = jnp.max(s, axis=0, keepdims=True)
                                pt = jnp.exp2(s - m_)
                                res.append((pt, m_, jnp.sum(pt, axis=0, keepdims=True)))
                            C[("p", b, g, p)] = res
                    elif op == "pv" and g_of(step) == 1 and c != 0:
                        _, b, g, ps = step[:4]
                        split = step[4] if len(step) > 4 else 1
                        need(*[("v", b, p, t) for p in ps for t in range(2)])
                        zero = jnp.zeros((64, 128), f32)
                        for p in ps:
                            res = C[("p", b, g, p)]
                            rows = pl.ds(b * 256 + p * 128, 128)
                            oo = []
                            for u in range(2):
                                js = qb_keys(u)
                                pt = res[u][0]
                                if len(js) == 2:
                                    assert js == [0, 3]
                                    vv = jnp.where(lane128, vtb[rows, 0:128], vtb[rows, 128:256])
                                else:
                                    j = js[0]
                                    vv = vtb[rows, pl.ds((j // 2) * 128, 128)]
                                    pt = jnp.concatenate([pt, zero] if j % 2 == 0 else [zero, pt], axis=0)
                                ptb = pt.astype(bf16)
                                if split > 1:
                                    oo.append([jnp.dot(vv[h * 64:(h + 1) * 64].astype(bf16), ptb, preferred_element_type=f32)
                                               for h in range(2)])
                                else:
                                    o = jnp.dot(vv.astype(bf16), ptb, preferred_element_type=f32)
                                    oo.append([o[0:64], o[64:128]])
                            l1 = lane64[0:1]
                            for h in range(2):
                                a_, b_ = (0, 1) if h == 0 else (1, 0)
                                vals = [jnp.where(lane64, oo[a_][h], oo[b_][h]),
                                        jnp.where(l1, res[a_][1], res[b_][1]), jnp.where(l1, res[a_][2], res[b_][2])]
                                if h == 1:
                                    C[("swapped", b, g, p)] = vals
                                else:
                                    put((b, g, p), h, frozenset([c]), *vals)
                    elif op == "s":
                        _, b, g, ps = step[:4]
                        split = step[4] if len(step) > 4 else 1
                        kbs = _key_blocks(c, g)
                        wait_msgs([(m, 0) for p in ps for m in kv_in((b, g, p))])
                        ss_ = {}
                        for p in ps:
                            pc = (b, g, p)
                            qm = C[("q", b, g, p)]
                            kall = jnp.concatenate([C[("k", b, p, j)] for j, _ in kbs], axis=0)
                            nk = kall.shape[0] // split
                            s = jnp.concatenate([
                                lax.dot_general(kall[i * nk:(i + 1) * nk].astype(bf16), qm, NT, preferred_element_type=f32)
                                for i in range(split)], axis=0)
                            blocks = []
                            for n_, (j, a) in enumerate(kbs):
                                sb = s[n_ * 64:(n_ + 1) * 64]
                                if not a[0]:
                                    sb = jnp.where(lane256, NEG, sb)
                                if not a[1]:
                                    sb = jnp.where(lane256, sb, NEG)
                                blocks.append(sb)
                            for m in kv_in(pc):
                                blocks.append(lax.dot_general(rbuf[pl.ds(rslot[m] * 64, nblk(m) * 64)], qm, NT,
                                                              preferred_element_type=f32))
                            ss_[p] = blocks
                        for p in ps:
                            s = jnp.concatenate(ss_[p], axis=0)
                            m_ = jnp.max(s, axis=0, keepdims=True)
                            pt = jnp.exp2(s - m_)
                            l = jnp.sum(pt, axis=0, keepdims=True)
                            C[("p", b, g, p)] = (pt, m_, l)
                    elif op == "pv":
                        _, b, g, ps = step[:4]
                        js = [j for j, _ in _key_blocks(c, g)]
                        need(*[("v", b, p, j // 2) for p in ps for j in js])
                        wait_msgs([(m, 1) for p in ps for m in kv_in((b, g, p))])
                        zero = jnp.zeros((64, 128), f32)
                        for p in ps:
                            pc = (b, g, p)
                            pt, m_, l = C[("p", b, g, p)]
                            for h in range(2):
                                r0 = b * 256 + p * 128 + h * 64
                                cols = slice(h * 128, (h + 1) * 128)
                                rows = {j: pt[n_ * 64:(n_ + 1) * 64, cols] for n_, j in enumerate(js)}
                                terms = []
                                if set(js) in ({0, 3}, {1, 2}):
                                    ev = [j for j in js if j % 2 == 0][0]
                                    od = [j for j in js if j % 2 == 1][0]
                                    vsel = jnp.where(lane64, vtb[pl.ds(r0, 64), pl.ds((ev // 2) * 128, 128)],
                                                     vtb[pl.ds(r0, 64), pl.ds((od // 2) * 128, 128)])
                                    terms.append((vsel.astype(bf16), jnp.concatenate([rows[ev], rows[od]], axis=0)))
                                else:
                                    for t in range(2):
                                        if 2 * t in rows or 2 * t + 1 in rows:
                                            terms.append((vtb[pl.ds(r0, 64), pl.ds(t * 128, 128)].astype(bf16),
                                                          jnp.concatenate([rows.get(2 * t, zero), rows.get(2 * t + 1, zero)], axis=0)))
                                off = len(js) * 64
                                for m in kv_in(pc):
                                    n = nblk(m)
                                    pr = pt[off:off + n * 64, cols]
                                    off += n * 64
                                    if n == 1:
                                        terms.append((rbuf[pl.ds((rslot[m] + 1) * 64, 64)],
                                                      jnp.concatenate([pr, zero] if h == 0 else [zero, pr], axis=0)))
                                    else:
                                        terms.append((rbuf[pl.ds((rslot[m] + 2 + h) * 64, 64)], pr))
                                o = add([jnp.dot(vv, pp.astype(bf16), preferred_element_type=f32) for vv, pp in terms])
                                ct = frozenset([c] + [m[1] for m in kv_in(pc)])
                                put(pc, h, ct, o, m_[:, cols], l[:, cols])
                    elif op == "recv":
                        lst = []
                        for b, g, p, src, hs in step[1]:
                            pc = (b, g, p)
                            m = [m for m in msgs if m[0] == pc and m[1] == src and m[2] == c and not is_kv(m)
                                 and any(("got", m, h) not in C for h in range(nparts(m)))][0]
                            if hs == "all":
                                hs = range(nparts(m))
                            lst += [(m, h) for h in hs]
                        wait_msgs(lst)
                        for m, h in lst:
                            if m[3] == ALL:
                                if all(("got", m, k) in C for k in range(2)):
                                    final.add(m[0])
                            else:
                                nr = 128 // nsub(m[0])
                                rs, hd = rslot[m], h * nr // 64
                                have[m[0] + (h,)][m[3]] = (rbuf[pl.ds(rs * 64 + h * nr, nr)].astype(f32),
                                                           rstat[rs + hd, 0:1], rstat[rs + hd, 1:2])
                    elif op == "flush":
                        for pc in step[1]:
                            flush(pc)
                        go()
                    elif op == "flushh":
                        for hd in range(2):
                            for pc in step[1]:
                                flush(pc, do_final=False, head=hd)
                            go()
                    elif op == "roll":
                        for pc in step[1]:
                            put(pc, 1, frozenset([c]), *[pltpu.roll(v, 64, 1) for v in C.pop(("swapped",) + pc)])
                    elif op == "stage":
                        for pc in step[1]:
                            flush(pc)
                    elif op == "fwd":
                        for pc in step[1]:
                            flush(pc, do_final=False)
                        go()
                    elif op == "go":
                        go()
                    elif op == "fence":
                        pl.semaphore_signal(rdy.at[c], inc=1)
                        pl.semaphore_wait(rdy.at[c], 1)
                    elif op == "drain":
                        n = len(started) - step[1]
                        for dsc in started[:n]:
                            dsc.wait_send()
                        del started[:n]
                    elif op == "wo":
                        need(("o",))
                        C["wo"] = [wob[0:128, :].astype(bf16), wob[128:256, :].astype(bf16)]
                        C["woh"] = {h: wob[h * 64:(h + 1) * 64, :].astype(bf16) for h in step[1:]}
                    elif op == "out" or op == "outh":
                        if op == "out":
                            _, b, g, ps = step
                            assert all((b, g, p) in final for p in ps), (c, step)
                            jobs = {(b, g): [(jnp.dot(fin[PID[(b, g, p)]], C["wo"][p], preferred_element_type=f32), 2)
                                             for p in ps]}
                        else:
                            jobs = {}
                            ts = []
                            for b, g, p, h in step[1]:
                                k = nsub((b, g, p)) // 2
                                o = []
                                for u in range(h * k, (h + 1) * k):
                                    parts = get((b, g, p, u), ALL)
                                    mm, a, l = merge(parts)
                                    inv = 1.0 / l
                                    o.append(add([(ai * inv) * pt[0] for ai, pt in zip(a, parts)]))
                                ts.append(jnp.concatenate(o, axis=0).T.astype(bf16))
                            for (b, g, p, h), t in zip(step[1], ts):
                                y = jnp.dot(t, C["woh"][2 * p + h], preferred_element_type=f32)
                                jobs.setdefault((b, g), []).append((y, 1))
                        for (b, g), terms in jobs.items():
                            if ("acc", b, g) in C:
                                terms = terms + [C.pop(("acc", b, g))]
                            o, n = add([t for t, _ in terms]), sum(n for _, n in terms)
                            if n < 4:
                                C[("acc", b, g)] = (o, n)
                                continue
                            if g == 0:
                                out_ref[b, 0:64, :] = o[0:64]
                                out_ref[b, 192:256, :] = o[64:128]
                            else:
                                out_ref[b, 64:192, :] = o
                            C[("done", b, g)] = True
                    else:
                        raise ValueError(step)
                assert not queue
                miss = [(m, h) for m in msgs for h in range(nparts(m)) if m[1] == c and (m, h) not in sent]
                assert not miss, (c, miss)
                miss = [(m, h) for m in msgs for h in range(nparts(m)) if m[2] == c and ("got", m, h) not in C]
                assert not miss, (c, miss)
                assert all(v[1] for v in loads.values()), (c, [k for k, v in loads.items() if not v[1]])
                assert all(("done", b, g) in C for b in range(2) for g in range(2)), c
                for d in ((1, 2, 3) if c == 0 else (2,) if c != 2 else ()):
                    know(d)
                with scope("Rend"):
                    for dsc in started:
                        dsc.wait_send()
                    if scopes:
                        pl.delay(1)

            for c in range(N_DEV):
                pl.when(my == c)(functools.partial(program, c))

        return pl.pallas_call(
            body,
            out_shape=jax.ShapeDtypeStruct((B, SQ, DM), f32),
            in_specs=[pl.BlockSpec(memory_space=pl.ANY)] * 5,
            out_specs=pl.BlockSpec(memory_space=pltpu.VMEM),
            scratch_shapes=[
                pltpu.VMEM((4, 128, DM), f32), pltpu.VMEM((DM, 256), f32),
                pltpu.VMEM((512, 256), f32), pltpu.VMEM((512, 256), f32), pltpu.VMEM((256, DM), f32),
                pltpu.VMEM((nss * 64, 128), bf16), pltpu.VMEM((nss, 2, 128), f32),
                pltpu.VMEM((nrs * 64, 128), bf16), pltpu.VMEM((nrs, 2, 128), f32),
                pltpu.VMEM((8, 128, 128), bf16),
                pltpu.SemaphoreType.DMA((32,)),
                pltpu.SemaphoreType.DMA((NSS,)), pltpu.SemaphoreType.DMA((NRS,)),
                pltpu.SemaphoreType.REGULAR((4,)),
            ],
            compiler_params=pltpu.CompilerParams(collective_id=0, disable_bounds_checks=True,
                                                 disable_semaphore_checks=True),
        )(x2, Wq, kt, vt, Wo)

    return kernel


P01 = (0, 1)
H01 = "all"
def plan():
    scheme = {}
    for p in range(2):
        scheme[(0,0,p)] = path(3,0,1,2)
        scheme[(1,0,p)] = path(2,3,0,1)
        scheme[(0,1,p)] = path(0,1,2,3,fa=0,fd=1)
        scheme[(1,1,p)] = path(1,2,3,0,fa=1,fd=0)
    fwd = {2: {(b,0,p) for b in range(2) for p in range(2)}, 1: {(1,0,0),(1,0,1)}, 3: {(0,0,0),(0,0,1)}}
    loads = {}; steps = {}
    for c, f in ((1, 1), (3, 0)):
        s = 1 - f
        if c == 1:
            l0 = [("k",(f,),(0,),P01), ("w",0), ("x",f,1), ("v",(f,),(0,),P01)]
            s0 = [("kprep",[(f,0,P01)]), ("kvK",[(f,0)]), ("go",), ("wq",(0,)), ("q",f,1,(0,)),
                  ("kvV",[(f,0)]), ("go",), ("s",f,1,(0,),2),
                  ("kprep",[(f,1,P01)]), ("pv",f,1,(0,),2), ("kvK",[(f,1)]), ("flush",[(f,1,0)])]
        else:
            l0 = [("v",(f,),(0,),P01), ("k",(f,),(0,),P01), ("w",0), ("x",f,1)]
            s0 = [("kvV",[(f,0)]), ("go",), ("kprep",[(f,0,P01)]), ("kvK",[(f,0)]), ("go",), ("wq",(0,)), ("q",f,1,(0,)),
                  ("kprep",[(f,1,P01)]), ("s",f,1,(0,),2), ("kvK",[(f,1)]), ("go",), ("fence",),
                  ("pv",f,1,(0,),2), ("flush",[(f,1,0)])]
        loads[c] = l0 + [("k",(f,),(1,),P01), ("w",1), ("v",(f,),(1,),P01),
                    ("k",(s,),(0,),P01), ("x",s,0), ("v",(s,),(0,),P01), ("k",(s,),(1,),P01), ("x",s,1), ("v",(s,),(1,),P01), ("o",)]
        steps[c] = s0 + [
                    ("wq",(1,)), ("roll",[(f,1,0)]), ("q",f,1,(1,)), ("flush",[(f,1,0)]),
                    ("kvV",[(f,1)]), ("s",f,1,(1,),2), ("go",),
                    ("kprep",[(s,0,P01)]), ("pv",f,1,(1,),2), ("flush",[(f,1,1)]),
                    ("xc",s,0), ("roll",[(f,1,1)]), ("q",s,0,(0,)), ("flush",[(f,1,1)]),
                    ("kvw",[(s,0,0)]), ("s",s,0,(0,)), ("q",s,0,(1,)),
                    ("kvw",[(s,0,1)]), ("kprep",[(s,1,P01)]), ("pv",s,0,(0,)), ("flush",[(s,0,0)]),
                    ("kvw",[(s,1,0)]), ("xc",s,1), ("s",s,0,(1,)), ("q",s,1,P01),
                    ("kvw",[(s,1,1)]), ("need",("v",s,1,0)), ("pv",s,0,(1,)), ("s",s,1,P01), ("flush",[(s,0,1)]),
                    ("recv",[(s,1,0,0,H01),(s,1,1,0,H01)]), ("pv",s,1,P01), ("flush",[(s,1,0)]), ("roll",[(s,1,0),(s,1,1)]), ("flush",[(s,1,0),(s,1,1)]),
                    ("wo",), ("drain",22),
                    ("recv",[(s,1,0,2,(0,1))]), ("fwd",[(s,1,0)]), ("recv",[(s,1,0,2,(2,))]), ("fwd",[(s,1,0)]), ("recv",[(s,1,0,2,(3,))]), ("fwd",[(s,1,0)]),
                    ("recv",[(s,1,1,2,(0,))]), ("fwd",[(s,1,1)]), ("recv",[(s,1,1,2,(1,))]), ("fwd",[(s,1,1)]),
                    ("recv",[(s,1,1,2,(2,))]), ("fwd",[(s,1,1)]), ("recv",[(s,1,1,2,(3,))]), ("fwd",[(s,1,1)]),
                    ("recv",[(s,0,0,0,H01)]), ("flush",[(s,0,0),(s,1,0),(s,1,1)]), ("recv",[(s,0,1,0,H01)]), ("flush",[(s,0,1)]),
                    ("out",s,1,P01), ("out",s,0,P01), ("drain",0),
                    ("recv",[(f,0,0,0,H01),(f,0,1,0,H01)]), ("out",f,0,P01),
                    ("recv",[(f,1,0,2,H01)]), ("out",f,1,(0,)), ("recv",[(f,1,1,2,H01)]), ("out",f,1,(1,))]
    loads[0] = [("w",0), ("x",0,1), ("x",1,1), ("k",(0,),(0,),P01), ("k",(1,),(0,),P01), ("v",(0,),(0,),P01), ("v",(1,),(0,),P01),
                ("w",1), ("k",(0,),(1,),P01), ("k",(1,),(1,),P01), ("v",(0,),(1,),P01), ("v",(1,),(1,),P01), ("x",1,0), ("x",0,0), ("o",)]
    steps[0] = [("wq",(0,)), ("q",0,1,(0,)), ("q",1,1,(0,)),
                ("kprep",[(0,0,P01),(1,0,P01)]), ("s",0,1,(0,)), ("s",1,1,(0,)),
                ("need",("v",1,0,0)), ("pv",0,1,(0,)), ("pv",1,1,(0,)), ("flush",[(0,1,0),(1,1,0)]),
                ("wq",(1,)), ("q",0,1,(1,)), ("q",1,1,(1,)),
                ("kprep",[(0,1,P01),(1,1,P01)]), ("s",0,1,(1,)), ("s",1,1,(1,)),
                ("need",("v",1,1,0)), ("pv",0,1,(1,)), ("pv",1,1,(1,)), ("flush",[(0,1,1),(1,1,1)]),
                ("q",1,0,P01),
                ("kvw",[(1,0,0)]), ("xc",0,0), ("s",1,0,(0,)), ("q",0,0,P01),
                ("kvw",[(1,0,1),(0,0,0),(0,0,1)]), ("pv",1,0,(0,)), ("s",0,0,(0,)), ("flush",[(1,0,0)]),
                ("kvw",[(1,1,0)]), ("wo",), ("pv",0,0,(0,)), ("s",1,0,(1,)), ("flush",[(0,0,0)]),
                ("kvw",[(1,1,1),(0,1,0)]), ("pv",1,0,(1,)), ("s",0,0,(1,)), ("flush",[(1,0,1)]),
                ("pv",0,0,(1,)), ("flush",[(0,0,1)]), ("drain",12),
                ("recv",[(0,0,0,1,H01),(1,0,0,3,H01)]), ("flush",[(0,0,0),(1,0,0)]), ("out",0,0,(0,)), ("out",1,0,(0,)),
                ("recv",[(0,0,1,1,H01),(1,0,1,3,H01)]), ("flush",[(0,0,1),(1,0,1)]), ("out",0,0,(1,)), ("out",1,0,(1,)),
                ("recv",[(0,1,0,1,H01),(1,1,0,3,H01)]), ("flush",[(0,1,0),(1,1,0)]), ("out",0,1,(0,)), ("out",1,1,(0,)), ("drain",0),
                ("recv",[(0,1,1,1,H01),(1,1,1,3,H01)]), ("flush",[(0,1,1),(1,1,1)]), ("out",0,1,(1,)), ("out",1,1,(1,))]
    loads[2] = [("k",(1,),(0,),(0,)), ("k",(0,),(0,),(0,)), ("v",(1,),(0,),(0,)), ("v",(0,),(0,),(0,)),
                ("k",(0,),(1,),(0,)), ("k",(1,),(1,),(0,)), ("v",(0,),(1,),(0,)), ("v",(1,),(1,),(0,)),
                ("w",0), ("x",0,1), ("x",1,1), ("k",(0,),(0,),(1,)), ("k",(1,),(0,),(1,)), ("v",(0,),(0,),(1,)), ("v",(1,),(0,),(1,)),
                ("w",1), ("k",(0,),(1,),(1,)), ("k",(1,),(1,),(1,)), ("v",(0,),(1,),(1,)), ("v",(1,),(1,),(1,)), ("o",)]
    steps[2] = [("kprep",[(0,0,(0,)),(1,0,(0,))]), ("kvK",[(0,0),(1,0)]), ("go",),
                ("kprep",[(0,1,(0,)),(1,1,(0,))]), ("kvV",[(0,0),(1,0)]), ("kvK",[(0,1),(1,1)]), ("go",),
                ("kvV",[(0,1),(1,1)]), ("go",),
                ("wq",(0,)), ("q",0,1,(0,)), ("q",1,1,(0,)),
                ("kprep",[(0,0,(1,)),(1,0,(1,))]), ("s",0,1,(0,)), ("s",1,1,(0,)),
                ("need",("v",1,0,1)), ("pv",0,1,(0,)), ("pv",1,1,(0,)),
                ("recv",[(0,1,0,3,(0,1)),(1,1,0,1,(0,1))]), ("fwd",[(0,1,0),(1,1,0)]),
                ("kprep",[(0,1,(1,)),(1,1,(1,))]), ("roll",[(0,1,0),(1,1,0)]), ("wq",(1,)), ("q",0,1,(1,)), ("q",1,1,(1,)),
                ("recv",[(0,1,0,3,(2,3)),(1,1,0,1,(2,3))]), ("fwd",[(0,1,0),(1,1,0)]), ("need",("v",1,1,1)),
                ("s",0,1,(1,)), ("s",1,1,(1,)),
                ("recv",[(0,1,1,3,(0,1)),(1,1,1,1,(0,1))]), ("pv",0,1,(1,)), ("pv",1,1,(1,)), ("fwd",[(0,1,1),(1,1,1)]), ("roll",[(0,1,1),(1,1,1)]),
                ("recv",[(0,1,1,3,(2,3)),(1,1,1,1,(2,3))]), ("fwd",[(0,1,1),(1,1,1)]),
                ("wo",),
                ("recv",[(0,1,0,1,H01),(1,1,0,3,H01)]), ("flush",[(0,1,0),(1,1,0)]),
                ("recv",[(0,1,1,1,H01),(1,1,1,3,H01)]), ("flush",[(0,1,1),(1,1,1)]),
                ("out",0,1,P01), ("out",1,1,P01), ("drain",0),
                ("recv",[(1,0,0,3,H01),(1,0,1,3,H01)]), ("out",1,0,P01),
                ("recv",[(0,0,0,1,H01),(0,0,1,1,H01)]), ("out",0,0,P01)]
    return scheme, fwd, loads, steps, {(0,1,0),(1,1,0),(0,1,1),(1,1,1)}


def pallas_dist_sparse_attn_blocksparse_kvseq_b2_sq256_skv256_hq4_dh64_kernel(x, Wq, K_ext, V_ext, Wo):
    return make_kernel(*plan())(x, Wq, K_ext, V_ext, Wo)
```

```python
import contextlib
import functools
import jax
import jax.numpy as jnp
from jax import lax
from jax.experimental import pallas as pl
from jax.experimental.pallas import tpu as pltpu

N_DEV = 4
B, SQ, DM, H, DH = 2, 256, 512, 4, 64
NEG = -1e9
LOG2E = 1.4426950408889634
f32 = jnp.float32
bf16 = jnp.bfloat16
MESH = pl.DeviceIdType.MESH
ALL = frozenset(range(4))
GROUP_QB = {0: (0, 3), 1: (1, 2)}
NT = (((1,), (1,)), ((), ()))
add = lambda xs: functools.reduce(lambda u, v: u + v, xs)


def _allowed(qb, kb):
    return qb == kb or kb == 0 or (qb + kb) % 3 == 0


def _key_blocks(chip, g):
    out = []
    for j in range(4):
        kb = 4 * chip + j
        a = tuple(_allowed(qb, kb) for qb in GROUP_QB[g])
        if any(a):
            out.append((j, a))
    return out


PIECES = [(b, g, p) for b in range(2) for g in range(2) for p in range(2)]
PID = {pc: i for i, pc in enumerate(PIECES)}


def path(a, b, c, d, fa=1, fd=1):
    F = frozenset
    return [(a, b, F([a])), (d, c, F([d])), (b, c, F([a, b])), (c, b, F([c, d])),
            (b, a, ALL if fa else F([b, c, d])), (c, d, ALL if fd else F([a, b, c]))]


def make_kernel(scheme, fwd, loads_order, steps, fine=(), qdst=None, scopes=False):
    msgs = [(pc, s, d, ct) for pc in PIECES for (s, d, ct) in scheme[pc]]
    MID = {m: i for i, m in enumerate(msgs)}

    def nsub(pc):
        return 4 if pc in fine else 2

    def nparts(m):
        if is_kv(m):
            return 1 + nblk(m)
        return 2 if m[3] == ALL else nsub(m[0])

    def is_kv(m):
        return len(m[3]) == 1 and m[0] in fwd.get(m[1], ())

    def nblk(m):
        return len(_key_blocks(m[1], m[0][1]))

    rslot, cnt = {}, [0] * 4
    for m in msgs:
        if m[3] != ALL:
            rslot[m] = cnt[m[2]]
            cnt[m[2]] += 2 * (nblk(m) if is_kv(m) else 1)
    nrs = max(cnt)
    sslot, cnt = {}, [0] * 4
    for m in msgs:
        pc, s, d, ct = m
        if ct != ALL and (pc, s, ct) not in sslot:
            sslot[(pc, s, ct)] = cnt[s]
            cnt[s] += 2 * (nblk(m) if is_kv(m) else 1)
    nss = max(cnt)
    ssem_id, rsem_id = {}, {}
    sc, rc_ = [0] * 4, [0] * 4
    for m in msgs:
        for u in range(nparts(m)):
            for kind in range(2):
                if kind == 1 and (m[3] == ALL or is_kv(m) or u > 0):
                    continue
                ssem_id[(m, u, kind)] = sc[m[1]]
                rsem_id[(m, u, kind)] = rc_[m[2]]
                sc[m[1]] += 1
                rc_[m[2]] += 1
    NSS, NRS = max(sc), max(rc_)

    def kernel(x, Wq, K_ext, V_ext, Wo):
        kt = jnp.transpose(K_ext, (0, 2, 3, 1)).reshape(B * H * DH, SQ)
        vt = jnp.transpose(V_ext, (0, 2, 3, 1)).reshape(B * H * DH, SQ)
        x2 = x.reshape(B * SQ, DM)

        def body(x_hbm, wq_hbm, kt_hbm, vt_hbm, wo_hbm, out_ref,
                 xb, wqb, ktb, vtb, wob, sbuf, sstat, rbuf, rstat, fin, qbuf,
                 lsem, s_sem, r_sem, qs_sem, qr_sem, rdy):
            my = lax.axis_index("i")
            bar = pltpu.get_barrier_semaphore()

            def program(c):
                nsc = [0]

                def scope(name):
                    nsc[0] += 1
                    on = scopes and (scopes is True or name[0] in scopes)
                    return jax.named_scope(f"s{nsc[0]:02d}_{name}") if on else contextlib.nullcontext()

                loads = {}

                def ld(key, src, dst):
                    cp = pltpu.make_async_copy(src, dst, lsem.at[len(loads)])
                    cp.start()
                    loads[key] = [cp, False]

                alias = {}
                for ck in loads_order[c]:
                    kind = ck[0]
                    if kind == "w":
                        if len(ck) == 1:
                            ld(ck, wq_hbm, wqb)
                            alias[("w", 0)] = alias[("w", 1)] = [ck]
                        else:
                            sl = pl.ds(ck[1] * 128, 128)
                            ld(ck, wq_hbm.at[:, sl], wqb.at[:, sl])
                            alias[ck] = [ck]
                    elif kind == "x":
                        _, b, g = ck
                        if g == 0:
                            ld(ck + (0,), x_hbm.at[pl.ds(b * 256, 64)], xb.at[b * 2, pl.ds(0, 64)])
                            ld(ck + (1,), x_hbm.at[pl.ds(b * 256 + 192, 64)], xb.at[b * 2, pl.ds(64, 64)])
                            alias[ck] = [ck + (0,), ck + (1,)]
                        else:
                            ld(ck, x_hbm.at[pl.ds(b * 256 + 64, 128)], xb.at[b * 2 + 1])
                            alias[ck] = [ck]
                    elif kind == "xh":
                        _, b, u = ck
                        ld(ck, x_hbm.at[pl.ds(b * 256 + 64 + u * 64, 64)], xb.at[b * 2 + 1, pl.ds(u * 64, 64)])
                        alias[ck] = [ck]
                    elif kind == "vh":
                        _, b, p, h = ck
                        rows = pl.ds(b * 256 + p * 128 + h * 64, 64)
                        ld(ck, vt_hbm.at[rows], vtb.at[rows])
                        alias[ck] = [ck]
                        for t in range(2):
                            alias.setdefault(("v", b, p, t), []).append(ck)
                    elif kind in ("k", "v"):
                        _, bs, ps, ts = ck
                        src, dst = (kt_hbm, ktb) if kind == "k" else (vt_hbm, vtb)
                        r0 = bs[0] * 256 + ps[0] * 128
                        nr = (256 * len(bs)) if len(ps) == 2 else 128
                        assert len(ps) == 2 or len(bs) == 1
                        rows = pl.ds(r0, nr)
                        if len(ts) == 2:
                            ld(ck, src.at[rows], dst.at[rows])
                        else:
                            cols = pl.ds(ts[0] * 128, 128)
                            ld(ck, src.at[rows, cols], dst.at[rows, cols])
                        for b in bs:
                            for p in ps:
                                for t in ts:
                                    alias[(kind, b, p, t)] = [ck]
                    elif kind == "o":
                        ld(ck, wo_hbm, wob)
                        alias[ck] = [ck]

                known = set()
                if c == 0:
                    for d in (1, 3):
                        pl.semaphore_signal(bar, inc=1, device_id=(d,), device_id_type=MESH)
                elif c in (1, 3):
                    pl.semaphore_wait(bar, 1)
                    known.add(0)
                    pl.semaphore_signal(bar, inc=1, device_id=(2,), device_id_type=MESH)
                    pl.semaphore_signal(rdy.at[c], inc=1, device_id=(0,), device_id_type=MESH)
                else:
                    pl.semaphore_wait(bar, 2)
                    known.update((0, 1, 3))
                    for d in (1, 3, 0):
                        pl.semaphore_signal(rdy.at[2], inc=1, device_id=(d,), device_id_type=MESH)

                def know(d):
                    if d in known:
                        return
                    if c in (1, 3) and d in (1, 3):
                        d = 2
                    pl.semaphore_wait(rdy.at[d], 1)
                    known.add(d)
                    if d == 2:
                        known.update((1, 3) if c != 0 else ())

                def need(*keys):
                    order = list(loads)
                    last = max(order.index(k) for key in keys for k in alias[key])
                    todo = [k for k in order[:last + 1] if not loads[k][1]]
                    if todo:
                        with scope("L" + "".join(map(str, todo[-1])).replace(" ", "").replace(",", "").replace("(", "").replace(")", "")):
                            for k in todo:
                                loads[k][1] = True
                                loads[k][0].wait()

                lane64 = lax.broadcasted_iota(jnp.int32, (64, 128), 1) < 64
                lane128 = lax.broadcasted_iota(jnp.int32, (128, 128), 1) < 64
                lane256 = (lax.broadcasted_iota(jnp.int32, (64, 256), 1) % 128) < 64
                C = {}
                have = {pc + (u,): {} for pc in PIECES for u in range(nsub(pc))}
                lses = {pc: {} for pc in PIECES}
                final = set()
                sent = set()
                started = []
                queue = []

                def rc(src, dst, k, d):
                    return pltpu.make_async_remote_copy(src, dst, s_sem.at[ssem_id[k]], r_sem.at[rsem_id[k]],
                                                        device_id=(d,), device_id_type=MESH)

                def qdesc(b, p):
                    i = b * 2 + p
                    return pltpu.make_async_remote_copy(qbuf.at[i], qbuf.at[i], qs_sem.at[i], qr_sem.at[i],
                                                        device_id=(qdst[(b, p)],), device_id_type=MESH)

                def put(pc, h, ct, o):
                    k = nsub(pc) // 2
                    for i in range(k):
                        have[pc + (k * h + i,)][ct] = o[(64 // k) * i:(64 // k) * (i + 1)]

                def descs(m, h):
                    pc, s, d, ct = m
                    if ct == ALL:
                        r = fin.at[PID[pc], pl.ds(h * 64, 64)]
                        return [rc(r, r, (m, h, 0), d)]
                    ss, rs = sslot[(pc, s, ct)], rslot[m]
                    if is_kv(m):
                        n = nblk(m)
                        off, nr = (0, n * 64) if h == 0 else ((n + h - 1) * 64, 64)
                        return [rc(sbuf.at[pl.ds(ss * 64 + off, nr)], rbuf.at[pl.ds(rs * 64 + off, nr)], (m, h, 0), d)]
                    nr = 128 // nsub(pc)
                    out = []
                    if (m, h, 1) in ssem_id:
                        out.append(rc(sstat.at[ss // 2], rstat.at[rs // 2], (m, h, 1), d))
                    out.append(rc(sbuf.at[pl.ds(ss * 64 + h * nr, nr)], rbuf.at[pl.ds(rs * 64 + h * nr, nr)], (m, h, 0), d))
                    return out

                def tag(m, h):
                    return "".join(map(str, m[0])) + f"h{h}_" + ("F" if m[3] == ALL else "".join(map(str, sorted(m[3]))))

                def go():
                    if not queue:
                        return
                    for m, h in queue:
                        know(m[2])
                    with scope("S" + "+".join(tag(m, h) + f">{m[2]}" for m, h in queue)):
                        for m, h in queue:
                            for dsc in descs(m, h):
                                dsc.start()
                                started.append(dsc)
                    queue.clear()

                def cover(held, ct):
                    rem, parts = set(ct), []
                    for k in sorted(held, key=lambda k: -len(k)):
                        if k <= rem:
                            parts.append(k)
                            rem -= k
                    return parts if not rem else None

                def weights(pc, ct, parts):
                    key = ("wts", pc, ct, tuple(parts))
                    if key not in C:
                        ls = [lses[pc][k] for k in parts]
                        m = functools.reduce(jnp.maximum, ls)
                        a = [jnp.exp2(v - m) for v in ls]
                        s = add(a)
                        inv = 1.0 / s
                        C[key] = [ai * inv for ai in a]
                        lses[pc].setdefault(ct, m + jnp.log2(s))
                    return C[key]

                def merged(pc, u, ct):
                    hv = have[pc + (u,)]
                    if ct in hv:
                        return hv[ct]
                    parts = cover(hv, ct)
                    if parts is None:
                        return None
                    hd = u * 2 // nsub(pc)
                    w = weights(pc, ct, parts)
                    return add([wi[:, hd * 128:(hd + 1) * 128] * hv[k] for wi, k in zip(w, parts)])

                def flush(pc, do_final=True, head=None):
                    outs = [m for m in msgs if m[0] == pc and m[1] == c]
                    recv_final = any(m[0] == pc and m[2] == c and m[3] == ALL for m in msgs)
                    nr = 128 // nsub(pc)
                    for h in range(nsub(pc)):
                        if head is not None and h * nr // 64 != head:
                            continue
                        key = pc + (h,)
                        for m in outs:
                            ct = m[3]
                            if ct == ALL or is_kv(m) or (m, h) in sent:
                                continue
                            if ("stored", key, ct) not in C:
                                o = merged(pc, h, ct)
                                if o is None:
                                    continue
                                have[key][ct] = o
                                ss = sslot[(pc, c, ct)]
                                sbuf[pl.ds(ss * 64 + h * nr, nr)] = o.astype(bf16)
                                if h == 0:
                                    sstat[ss // 2] = lses[pc][ct]
                                C[("stored", key, ct)] = True
                            sent.add((m, h))
                            queue.append((m, h))
                    if do_final and pc not in final and not recv_final:
                        if all(cover(have[pc + (h,)], ALL) is not None for h in range(nsub(pc))):
                            o = [merged(pc, h, ALL) for h in range(nsub(pc))]
                            t = jnp.concatenate(o, axis=0).T
                            fin[PID[pc]] = t.astype(bf16)
                            final.add(pc)
                    if pc in final:
                        for m in outs:
                            for h in range(2):
                                if m[3] == ALL and (m, h) not in sent:
                                    sent.add((m, h))
                                    queue.append((m, h))

                def wait_msgs(lst):
                    lst = [(m, h) for m, h in lst if ("got", m, h) not in C]
                    if not lst:
                        return
                    with scope("R" + "+".join(tag(m, h) + f"<{m[1]}" for m, h in lst)):
                        for m, h in lst:
                            for dsc in descs(m, h):
                                dsc.wait_recv()
                            C[("got", m, h)] = True

                def g_of(step):
                    return step[2]

                def qb_keys(u):
                    return [j for j, a in _key_blocks(c, 1) if a[u]]

                def kv_in(pc):
                    return [m for m in msgs if m[0] == pc and m[2] == c and is_kv(m)]

                for step in steps[c]:
                    op = step[0]
                    if op == "need":
                        need(*step[1:])
                    elif op == "kvw":
                        wait_msgs([(m, u) for b, p, part in step[1] for m in kv_in((b, 0, p))
                                   for u in ([0] if part == 0 else range(1, nparts(m)))])
                    elif op == "kprep":
                        need(*[("k", b, p, t) for b, p, ts in step[1] for t in ts])
                        for b, p, ts in step[1]:
                            kk = ktb[pl.ds(b * 256 + p * 128, 128), pl.ds(ts[0] * 128, 128 * len(ts))].T
                            for n_, t in enumerate(ts):
                                for jj in range(2):
                                    C[("k", b, p, 2 * t + jj)] = kk[n_ * 128 + jj * 64: n_ * 128 + jj * 64 + 64]
                    elif op == "kvK" or op == "kvV":
                        js = [j for j, _ in _key_blocks(c, 0)]
                        n = len(js)
                        heads = step[2] if len(step) > 2 else (0, 1)
                        if op == "kvV":
                            if len(step) > 2:
                                need(*[("vh", b, p, h) for b, p in step[1] for h in heads])
                            else:
                                need(*[("v", b, p, j // 2) for b, p in step[1] for j in js])
                        for b, p in step[1]:
                            pc = (b, 0, p)
                            ss = sslot[(pc, c, frozenset([c]))]
                            if op == "kvK":
                                parts = [0]
                                for n_, j in enumerate(js):
                                    sbuf[pl.ds((ss + n_) * 64, 64)] = C[("k", b, p, j)].astype(bf16)
                            elif n == 1:
                                parts = [1]
                                j = js[0]
                                v = vtb[pl.ds(b * 256 + p * 128, 128), pl.ds((j // 2) * 128, 128)]
                                v0, v1 = v[0:64], v[64:128]
                                if j % 2 == 1:
                                    v0 = pltpu.roll(v0, 64, 1)
                                else:
                                    v1 = pltpu.roll(v1, 64, 1)
                                sbuf[pl.ds((ss + 1) * 64, 64)] = jnp.where(lane64, v0, v1).astype(bf16)
                            else:
                                assert js == [0, 3]
                                parts = [1 + h for h in heads]
                                for h in heads:
                                    rows = pl.ds(b * 256 + p * 128 + h * 64, 64)
                                    sbuf[pl.ds((ss + 2 + h) * 64, 64)] = jnp.where(
                                        lane64, vtb[rows, 0:128], vtb[rows, 128:256]).astype(bf16)
                            for m in msgs:
                                if m[0] == pc and m[1] == c and is_kv(m):
                                    for hh in parts:
                                        sent.add((m, hh))
                                        queue.append((m, hh))
                    elif op == "wq":
                        ps = step[1]
                        need(*[("w", p) for p in ps])
                        for p in ps:
                            C[("w", p)] = wqb[:, pl.ds(p * 128, 128)].astype(bf16)
                    elif op == "xc":
                        _, b, g = step
                        need(("x", b, g))
                        C[("x", b, g)] = xb[b * 2 + g].astype(bf16)
                    elif op == "q":
                        _, b, g, ps = step
                        if ("x", b, g) not in C:
                            need(("x", b, g))
                            C[("x", b, g)] = xb[b * 2 + g].astype(bf16)
                        for p in ps:
                            qp = jnp.dot(C[("x", b, g)], C[("w", p)], preferred_element_type=f32) * (0.125 * LOG2E)
                            C[("qraw", b, g, p)] = qp
                            q0, q1 = jnp.where(lane128, qp, 0.0), jnp.where(lane128, 0.0, qp)
                            if g == 0 or c == 0:
                                tiles = [q0, q1]
                            else:
                                tiles = None
                                C[("q", b, g, p)] = [jnp.concatenate([q0[0:64], q1[0:64]], axis=0).astype(bf16),
                                                     jnp.concatenate([q1[64:128], q0[64:128]], axis=0).astype(bf16)]
                            if tiles is not None:
                                C[("q", b, g, p)] = jnp.concatenate(tiles, axis=0).astype(bf16)
                    elif op == "qh":
                        _, b, u, ps = step
                        need(("xh", b, u))
                        xv = xb[b * 2 + 1, pl.ds(u * 64, 64)].astype(bf16)
                        for p in ps:
                            qp = jnp.dot(xv, C[("w", p)], preferred_element_type=f32) * (0.125 * LOG2E)
                            q0, q1 = jnp.where(lane64, qp, 0.0), jnp.where(lane64, 0.0, qp)
                            C.setdefault(("q", b, 1, p), [None, None])[u] = jnp.concatenate(
                                [q0, q1] if u == 0 else [q1, q0], axis=0).astype(bf16)
                    elif op == "qsend":
                        for b, p in step[1]:
                            qbuf[b * 2 + p] = C[("qraw", b, 0, p)].astype(bf16)
                        for b, p in step[1]:
                            know(qdst[(b, p)])
                        with scope("SQ"):
                            for b, p in step[1]:
                                dsc = qdesc(b, p)
                                dsc.start()
                                started.append(dsc)
                    elif op == "qrecv":
                        with scope("RQ" + "".join(f"{b}{p}" for b, p in step[1])):
                            for b, p in step[1]:
                                qdesc(b, p).wait_recv()
                        for b, p in step[1]:
                            qp = qbuf[b * 2 + p].astype(f32)
                            C[("q", b, 0, p)] = jnp.concatenate(
                                [jnp.where(lane128, qp, 0.0), jnp.where(lane128, 0.0, qp)], axis=0).astype(bf16)
                    elif op == "s" and g_of(step) == 1 and c != 0:
                        _, b, g, ps = step[:4]
                        split = step[4] if len(step) > 4 else 1
                        kbs = _key_blocks(c, g)
                        ss_ = {}
                        for p in ps:
                            for u in range(2):
                                js = qb_keys(u)
                                if split > 1:
                                    ss_[(p, u)] = jnp.concatenate([
                                        lax.dot_general(C[("k", b, p, j)].astype(bf16), C[("q", b, g, p)][u], NT,
                                                        preferred_element_type=f32) for j in js], axis=0)
                                else:
                                    kall = jnp.concatenate([C[("k", b, p, j)] for j in js], axis=0).astype(bf16)
                                    ss_[(p, u)] = lax.dot_general(kall, C[("q", b, g, p)][u], NT, preferred_element_type=f32)
                        for p in ps:
                            res = []
                            for u in range(2):
                                s = ss_[(p, u)]
                                m_ = jnp.max(s, axis=0, keepdims=True)
                                pt = jnp.exp2(s - m_)
                                l = jnp.sum(pt, axis=0, keepdims=True)
                                res.append((pt, 1.0 / l, m_ + jnp.log2(l)))
                            C[("p", b, g, p)] = res
                    elif op == "pv" and g_of(step) == 1 and c != 0:
                        _, b, g, ps = step[:4]
                        split = step[4] if len(step) > 4 else 1
                        need(*[("v", b, p, t) for p in ps for t in range(2)])
                        zero = jnp.zeros((64, 128), f32)
                        for p in ps:
                            res = C[("p", b, g, p)]
                            rows = pl.ds(b * 256 + p * 128, 128)
                            oo = []
                            for u in range(2):
                                js = qb_keys(u)
                                pt = res[u][0]
                                if len(js) == 2:
                                    assert js == [0, 3]
                                    vv = jnp.where(lane128, vtb[rows, 0:128], vtb[rows, 128:256])
                                else:
                                    j = js[0]
                                    vv = vtb[rows, pl.ds((j // 2) * 128, 128)]
                                    pt = jnp.concatenate([pt, zero] if j % 2 == 0 else [zero, pt], axis=0)
                                ptb = pt.astype(bf16)
                                if split > 1:
                                    oo.append([jnp.dot(vv[h * 64:(h + 1) * 64].astype(bf16), ptb, preferred_element_type=f32)
                                               for h in range(2)])
                                else:
                                    o = jnp.dot(vv.astype(bf16), ptb, preferred_element_type=f32)
                                    oo.append([o[0:64], o[64:128]])
                            l1 = lane64[0:1]
                            me = frozenset([c])
                            lses[(b, g, p)][me] = jnp.concatenate(
                                [jnp.where(l1, res[0][2], res[1][2]),
                                 pltpu.roll(jnp.where(l1, res[1][2], res[0][2]), 64, 1)], axis=1)
                            put((b, g, p), 0, me, jnp.where(lane64, oo[0][0], oo[1][0]) * jnp.where(l1, res[0][1], res[1][1]))
                            C[("swapped", b, g, p)] = (jnp.where(lane64, oo[1][1], oo[0][1])
                                                       * jnp.where(l1, res[1][1], res[0][1]))
                    elif op == "s":
                        _, b, g, ps = step[:4]
                        split = step[4] if len(step) > 4 else 1
                        kbs = _key_blocks(c, g)
                        wait_msgs([(m, 0) for p in ps for m in kv_in((b, g, p))])
                        ss_ = {}
                        for p in ps:
                            pc = (b, g, p)
                            qm = C[("q", b, g, p)]
                            kall = jnp.concatenate([C[("k", b, p, j)] for j, _ in kbs], axis=0)
                            nk = kall.shape[0] // split
                            s = jnp.concatenate([
                                lax.dot_general(kall[i * nk:(i + 1) * nk].astype(bf16), qm, NT, preferred_element_type=f32)
                                for i in range(split)], axis=0)
                            blocks = []
                            for n_, (j, a) in enumerate(kbs):
                                sb = s[n_ * 64:(n_ + 1) * 64]
                                if not a[0]:
                                    sb = jnp.where(lane256, NEG, sb)
                                if not a[1]:
                                    sb = jnp.where(lane256, sb, NEG)
                                blocks.append(sb)
                            for m in kv_in(pc):
                                blocks.append(lax.dot_general(rbuf[pl.ds(rslot[m] * 64, nblk(m) * 64)], qm, NT,
                                                              preferred_element_type=f32))
                            ss_[p] = blocks
                        for p in ps:
                            s = jnp.concatenate(ss_[p], axis=0)
                            m_ = jnp.max(s, axis=0, keepdims=True)
                            pt = jnp.exp2(s - m_)
                            l = jnp.sum(pt, axis=0, keepdims=True)
                            C[("p", b, g, p)] = (pt, 1.0 / l, m_ + jnp.log2(l))
                    elif op == "pv":
                        _, b, g, ps = step[:4]
                        js = [j for j, _ in _key_blocks(c, g)]
                        need(*[("v", b, p, j // 2) for p in ps for j in js])
                        wait_msgs([(m, u) for p in ps for m in kv_in((b, g, p)) for u in range(1, nparts(m))])
                        zero = jnp.zeros((64, 128), f32)
                        for p in ps:
                            pc = (b, g, p)
                            pt, inv, lse = C[("p", b, g, p)]
                            for h in range(2):
                                r0 = b * 256 + p * 128 + h * 64
                                cols = slice(h * 128, (h + 1) * 128)
                                rows = {j: pt[n_ * 64:(n_ + 1) * 64, cols] for n_, j in enumerate(js)}
                                terms = []
                                if set(js) in ({0, 3}, {1, 2}):
                                    ev = [j for j in js if j % 2 == 0][0]
                                    od = [j for j in js if j % 2 == 1][0]
                                    vsel = jnp.where(lane64, vtb[pl.ds(r0, 64), pl.ds((ev // 2) * 128, 128)],
                                                     vtb[pl.ds(r0, 64), pl.ds((od // 2) * 128, 128)])
                                    terms.append((vsel.astype(bf16), jnp.concatenate([rows[ev], rows[od]], axis=0)))
                                else:
                                    for t in range(2):
                                        if 2 * t in rows or 2 * t + 1 in rows:
                                            terms.append((vtb[pl.ds(r0, 64), pl.ds(t * 128, 128)].astype(bf16),
                                                          jnp.concatenate([rows.get(2 * t, zero), rows.get(2 * t + 1, zero)], axis=0)))
                                off = len(js) * 64
                                for m in kv_in(pc):
                                    n = nblk(m)
                                    pr = pt[off:off + n * 64, cols]
                                    off += n * 64
                                    if n == 1:
                                        terms.append((rbuf[pl.ds((rslot[m] + 1) * 64, 64)],
                                                      jnp.concatenate([pr, zero] if h == 0 else [zero, pr], axis=0)))
                                    else:
                                        terms.append((rbuf[pl.ds((rslot[m] + 2 + h) * 64, 64)], pr))
                                o = add([jnp.dot(vv, pp.astype(bf16), preferred_element_type=f32) for vv, pp in terms])
                                ct = frozenset([c] + [m[1] for m in kv_in(pc)])
                                put(pc, h, ct, o * inv[:, cols])
                                lses[pc][ct] = lse
                    elif op == "recv":
                        lst = []
                        for b, g, p, src, hs in step[1]:
                            pc = (b, g, p)
                            m = [m for m in msgs if m[0] == pc and m[1] == src and m[2] == c and not is_kv(m)
                                 and any(("got", m, h) not in C for h in range(nparts(m)))][0]
                            if hs == "all":
                                hs = range(nparts(m))
                            lst += [(m, h) for h in hs]
                        wait_msgs(lst)
                        for m, h in lst:
                            if m[3] == ALL:
                                if all(("got", m, k) in C for k in range(2)):
                                    final.add(m[0])
                            else:
                                nr = 128 // nsub(m[0])
                                rs = rslot[m]
                                have[m[0] + (h,)][m[3]] = rbuf[pl.ds(rs * 64 + h * nr, nr)].astype(f32)
                                if h == 0:
                                    lses[m[0]][m[3]] = rstat[rs // 2]
                    elif op == "flush":
                        for pc in step[1]:
                            flush(pc)
                        go()
                    elif op == "flushh":
                        for hd in range(2):
                            for pc in step[1]:
                                flush(pc, do_final=False, head=hd)
                            go()
                    elif op == "roll":
                        for pc in step[1]:
                            put(pc, 1, frozenset([c]), pltpu.roll(C.pop(("swapped",) + pc), 64, 1))
                    elif op == "stage":
                        for pc in step[1]:
                            flush(pc)
                    elif op == "fwd":
                        for pc in step[1]:
                            flush(pc, do_final=False)
                        go()
                    elif op == "go":
                        go()
                    elif op == "fence":
                        pl.semaphore_signal(rdy.at[c], inc=1)
                        pl.semaphore_wait(rdy.at[c], 1)
                    elif op == "drain":
                        n = len(started) - step[1]
                        for dsc in started[:n]:
                            dsc.wait_send()
                        del started[:n]
                    elif op == "wo":
                        need(("o",))
                        C["wo"] = [wob[0:128, :].astype(bf16), wob[128:256, :].astype(bf16)]
                        if len(step) > 1:
                            C["wop"] = [jnp.concatenate([wob[h * 64:(h + 1) * 64, :], wob[128 + h * 64:128 + (h + 1) * 64, :]],
                                                        axis=0).astype(bf16) for h in range(2)]
                    elif op in ("out", "outh", "outp"):
                        if op == "outp":
                            _, b, g, h = step
                            o = []
                            for p in range(2):
                                k = nsub((b, g, p)) // 2
                                for u in range(h * k, (h + 1) * k):
                                    o.append(merged((b, g, p), u, ALL))
                            t = jnp.concatenate(o, axis=0).T.astype(bf16)
                            jobs = {(b, g): [(jnp.dot(t, C["wop"][h], preferred_element_type=f32), 2)]}
                        elif op == "out":
                            _, b, g, ps = step
                            assert all((b, g, p) in final for p in ps), (c, step)
                            jobs = {(b, g): [(jnp.dot(fin[PID[(b, g, p)]], C["wo"][p], preferred_element_type=f32), 2)
                                             for p in ps]}
                        else:
                            jobs = {}
                            ts = []
                            for b, g, p, h in step[1]:
                                k = nsub((b, g, p)) // 2
                                o = []
                                for u in range(h * k, (h + 1) * k):
                                    o.append(merged((b, g, p), u, ALL))
                                ts.append(jnp.concatenate(o, axis=0).T.astype(bf16))
                            for (b, g, p, h), t in zip(step[1], ts):
                                y = jnp.dot(t, C["woh"][2 * p + h], preferred_element_type=f32)
                                jobs.setdefault((b, g), []).append((y, 1))
                        for (b, g), terms in jobs.items():
                            if ("acc", b, g) in C:
                                terms = terms + [C.pop(("acc", b, g))]
                            o, n = add([t for t, _ in terms]), sum(n for _, n in terms)
                            if n < 4:
                                C[("acc", b, g)] = (o, n)
                                continue
                            if g == 0:
                                out_ref[b, 0:64, :] = o[0:64]
                                out_ref[b, 192:256, :] = o[64:128]
                            else:
                                out_ref[b, 64:192, :] = o
                            C[("done", b, g)] = True
                    else:
                        raise ValueError(step)
                assert not queue
                miss = [(m, h) for m in msgs for h in range(nparts(m)) if m[1] == c and (m, h) not in sent]
                assert not miss, (c, miss)
                miss = [(m, h) for m in msgs for h in range(nparts(m)) if m[2] == c and ("got", m, h) not in C]
                assert not miss, (c, miss)
                assert all(v[1] for v in loads.values()), (c, [k for k, v in loads.items() if not v[1]])
                assert all(("done", b, g) in C for b in range(2) for g in range(2)), c
                for d in ((1, 2, 3) if c == 0 else (2,) if c != 2 else ()):
                    know(d)
                with scope("Rend"):
                    for dsc in started:
                        dsc.wait_send()
                    if scopes:
                        pl.delay(1)

            for c in range(N_DEV):
                pl.when(my == c)(functools.partial(program, c))

        return pl.pallas_call(
            body,
            out_shape=jax.ShapeDtypeStruct((B, SQ, DM), f32),
            in_specs=[pl.BlockSpec(memory_space=pl.ANY)] * 5,
            out_specs=pl.BlockSpec(memory_space=pltpu.VMEM),
            scratch_shapes=[
                pltpu.VMEM((4, 128, DM), f32), pltpu.VMEM((DM, 256), f32),
                pltpu.VMEM((512, 256), f32), pltpu.VMEM((512, 256), f32), pltpu.VMEM((256, DM), f32),
                pltpu.VMEM((nss * 64, 128), bf16), pltpu.VMEM((nss // 2, 1, 256), f32),
                pltpu.VMEM((nrs * 64, 128), bf16), pltpu.VMEM((nrs // 2, 1, 256), f32),
                pltpu.VMEM((8, 128, 128), bf16), pltpu.VMEM((4, 128, 128), bf16),
                pltpu.SemaphoreType.DMA((32,)),
                pltpu.SemaphoreType.DMA((NSS,)), pltpu.SemaphoreType.DMA((NRS,)),
                pltpu.SemaphoreType.DMA((4,)), pltpu.SemaphoreType.DMA((4,)),
                pltpu.SemaphoreType.REGULAR((4,)),
            ],
            compiler_params=pltpu.CompilerParams(collective_id=0, disable_bounds_checks=True,
                                                 disable_semaphore_checks=True),
        )(x2, Wq, kt, vt, Wo)

    return kernel


P01 = (0, 1)
H01 = "all"
def plan():
    scheme = {}
    for b in range(2):
        scheme[(b,0,0)] = path(3,0,1,2)
        scheme[(b,0,1)] = path(2,3,0,1)
        scheme[(b,1,0)] = path(0,1,2,3,fa=0,fd=1)
        scheme[(b,1,1)] = path(1,2,3,0,fa=1,fd=0)
    fwd = {2: {(b,0,p) for b in range(2) for p in range(2)}, 1: {(0,0,1),(1,0,1)}, 3: {(0,0,0),(1,0,0)}}
    qdst = {(b,p): (1 if p == 0 else 3) for b in range(2) for p in range(2)}
    fine = {(b,1,p) for b in range(2) for p in range(2)}
    loads = {}; steps = {}
    for c, f in ((1, 1), (3, 0)):
        s = 1 - f
        F, S = (f,), (s,)
        if c == 1:
            l0 = [("k",(0,),F,P01), ("w",f), ("x",0,1), ("v",(0,),F,P01), ("k",(1,),F,P01), ("x",1,1), ("v",(1,),F,P01)]
            s0 = [("kprep",[(0,f,P01)]), ("kvK",[(0,f)]), ("go",), ("wq",F), ("q",0,1,F), ("s",0,1,F,2),
                  ("kprep",[(1,f,P01)]), ("pv",0,1,F,2), ("flush",[(0,1,f)]), ("kvV",[(0,f)]), ("kvK",[(1,f)]), ("go",),
                  ("xc",1,1), ("roll",[(0,1,f)]), ("q",1,1,F), ("flush",[(0,1,f)]),
                  ("kvV",[(1,f)]), ("s",1,1,F,2), ("go",),
                  ("kprep",[(0,s,P01)]), ("pv",1,1,F,2), ("flush",[(1,1,f)])]
        else:
            l0 = [("vh",0,f,0), ("k",(0,),F,P01), ("w",f), ("x",0,1), ("vh",0,f,1), ("v",(1,),F,P01), ("x",1,1), ("k",(1,),F,P01)]
            s0 = [("kvV",[(0,f)],(0,)), ("go",), ("kprep",[(0,f,P01)]), ("kvK",[(0,f)]), ("go",), ("wq",F),
                  ("q",0,1,F), ("kvV",[(0,f)],(1,)), ("go",), ("fence",), ("s",0,1,F,2), ("pv",0,1,F,2), ("flush",[(0,1,f)]),
                  ("kvV",[(1,f)]), ("go",),
                  ("xc",1,1), ("roll",[(0,1,f)]), ("q",1,1,F), ("flush",[(0,1,f)]),
                  ("kprep",[(1,f,P01)]), ("s",1,1,F,2), ("kvK",[(1,f)]), ("go",),
                  ("kprep",[(0,s,P01)]), ("pv",1,1,F,2), ("flush",[(1,1,f)])]
        loads[c] = l0 + [("k",(0,),S,P01), ("w",s), ("v",(0,),S,P01), ("k",(1,),S,P01), ("v",(1,),S,P01), ("o",)]
        steps[c] = s0 + [
                    ("qrecv",[(0,s)]), ("roll",[(1,1,f)]), ("flush",[(1,1,f)]),
                    ("kvw",[(0,s,0)]), ("wq",S), ("s",0,0,S), ("q",0,1,S),
                    ("kvw",[(0,s,1)]), ("kprep",[(1,s,P01)]), ("pv",0,0,S), ("q",1,1,S), ("flush",[(0,0,s)]),
                    ("kvw",[(1,s,0)]), ("qrecv",[(1,s)]), ("need",("v",1,s,0)), ("s",1,0,S), ("s",0,1,S), ("s",1,1,S),
                    ("kvw",[(1,s,1)]), ("pv",1,0,S), ("pv",0,1,S), ("pv",1,1,S), ("flush",[(1,0,s)]), ("roll",[(0,1,s),(1,1,s)]),
                    ("recv",[(0,1,s,0,H01)]), ("flush",[(0,1,s)]),
                    ("wo",), ("drain",14),
                    ("recv",[(1,1,s,0,(0,1))]), ("fwd",[(1,1,s)]),
                    ("recv",[(0,1,s,2,(0,))]), ("fwd",[(0,1,s)]), ("recv",[(1,1,s,0,(2,3))]), ("fwd",[(1,1,s)]),
                    ("recv",[(0,1,s,2,(1,))]), ("fwd",[(0,1,s)]), ("recv",[(0,1,s,2,(2,))]), ("fwd",[(0,1,s)]), ("recv",[(0,1,s,2,(3,))]), ("fwd",[(0,1,s)]),
                    ("recv",[(1,1,s,2,(0,))]), ("fwd",[(1,1,s)]), ("recv",[(1,1,s,2,(1,))]), ("fwd",[(1,1,s)]),
                    ("recv",[(1,1,s,2,(2,))]), ("fwd",[(1,1,s)]), ("recv",[(1,1,s,2,(3,))]), ("fwd",[(1,1,s)]),
                    ("recv",[(0,0,s,0,H01)]), ("flush",[(0,0,s),(0,1,s),(1,1,s)]), ("recv",[(1,0,s,0,H01)]), ("flush",[(1,0,s)]),
                    ("out",0,1,S), ("out",1,1,S), ("out",0,0,S), ("out",1,0,S), ("drain",6),
                    ("recv",[(0,0,f,0,H01)]), ("out",0,0,F), ("recv",[(0,1,f,2,H01)]), ("out",0,1,F),
                    ("recv",[(1,0,f,0,H01)]), ("out",1,0,F), ("recv",[(1,1,f,2,H01)]), ("out",1,1,F)]
    loads[0] = [("w",), ("x",0,0), ("x",1,0), ("x",0,1), ("k",(0,),P01,P01), ("v",(0,),P01,P01),
                ("x",1,1), ("k",(1,),P01,P01), ("v",(1,),P01,P01), ("o",)]
    steps[0] = [("wq",P01), ("q",0,0,P01), ("xc",1,0), ("q",1,0,P01), ("qsend",[(0,0),(0,1),(1,0),(1,1)]),
                ("q",0,1,P01), ("kprep",[(0,0,P01),(0,1,P01)]), ("s",0,1,P01),
                ("pv",0,1,P01), ("flush",[(0,1,0),(0,1,1)]),
                ("q",1,1,P01), ("kprep",[(1,0,P01),(1,1,P01)]), ("s",1,1,P01),
                ("pv",1,1,P01), ("flush",[(1,1,0),(1,1,1)]),
                ("kvw",[(0,1,0),(0,0,0)]), ("s",0,0,P01),
                ("kvw",[(0,1,1),(0,0,1),(1,1,0)]), ("wo",1), ("pv",0,0,P01), ("s",1,0,(1,)), ("flush",[(0,0,1),(0,0,0)]),
                ("kvw",[(1,1,1)]), ("pv",1,0,(1,)), ("flush",[(1,0,1)]),
                ("kvw",[(1,0,0),(1,0,1)]), ("s",1,0,(0,),2), ("pv",1,0,(0,)), ("flush",[(1,0,0)]), ("drain",12),
                ("recv",[(0,0,0,1,H01),(0,0,1,3,H01)]), ("flush",[(0,0,0),(0,0,1)]), ("out",0,0,P01),
                ("recv",[(1,0,0,1,H01),(1,0,1,3,H01)]), ("flush",[(1,0,0),(1,0,1)]), ("drain",8),
                ("recv",[(0,1,0,1,(0,1)),(0,1,1,3,(0,1))]), ("out",1,0,(0,)), ("outp",0,1,0),
                ("recv",[(0,1,0,1,(2,3)),(0,1,1,3,(2,3))]), ("out",1,0,(1,)), ("outp",0,1,1),
                ("recv",[(1,1,0,1,(0,1)),(1,1,1,3,(0,1))]), ("outp",1,1,0), ("drain",0),
                ("recv",[(1,1,0,1,(2,3)),(1,1,1,3,(2,3))]), ("outp",1,1,1)]
    loads[2] = [("k",(0,),P01,(0,)), ("v",(0,),P01,(0,)), ("k",(1,),P01,(0,)), ("v",(1,),P01,(0,)),
                ("w",0), ("x",0,1), ("w",1), ("k",(0,),P01,(1,)), ("v",(0,),P01,(1,)),
                ("xh",1,0), ("xh",1,1), ("k",(1,),P01,(1,)), ("v",(1,),P01,(1,)), ("o",)]
    R = lambda b, u: ("recv",[(b,1,0,3,u),(b,1,1,1,u)])
    W = lambda b: ("fwd",[(b,1,0),(b,1,1)])
    RO = lambda b: ("roll",[(b,1,0),(b,1,1)])
    KP = ("kprep",[(1,0,(1,)),(1,1,(1,))])
    steps[2] = [("kprep",[(0,0,(0,)),(0,1,(0,))]), ("kvK",[(0,0),(0,1)]), ("go",),
                ("kprep",[(1,0,(0,)),(1,1,(0,))]), ("kvV",[(0,0),(0,1)]), ("kvK",[(1,0),(1,1)]), ("go",),
                ("kvV",[(1,0),(1,1)]), ("go",),
                ("wq",(0,)), ("q",0,1,(0,)), ("wq",(1,)), ("q",0,1,(1,)),
                ("kprep",[(0,0,(1,)),(0,1,(1,))]), ("s",0,1,P01),
                ("need",("xh",1,0)), R(0,(0,)), ("pv",0,1,P01), ("qh",1,0,P01), W(0), RO(0),
                R(0,(1,2)), W(0),
                KP, ("qh",1,1,P01), ("s",1,1,P01),
                R(0,(3,)), W(0),
                ("need",("v",1,1,1)), R(1,(0,)), ("pv",1,1,P01), W(1), RO(1),
                R(1,(1,2)), W(1), R(1,(3,)), W(1),
                ("wo",),
                ("recv",[(0,1,0,1,H01),(0,1,1,3,H01)]), ("flush",[(0,1,0),(0,1,1)]), ("out",0,1,P01),
                ("recv",[(1,1,0,1,H01),(1,1,1,3,H01)]), ("flush",[(1,1,0),(1,1,1)]), ("out",1,1,P01), ("drain",4),
                ("recv",[(0,0,0,1,H01),(0,0,1,3,H01)]), ("out",0,0,P01),
                ("recv",[(1,0,0,1,H01),(1,0,1,3,H01)]), ("out",1,0,P01)]
    return scheme, fwd, loads, steps, fine, qdst


def pallas_dist_sparse_attn_blocksparse_kvseq_b2_sq256_skv256_hq4_dh64_kernel(x, Wq, K_ext, V_ext, Wo):
    return make_kernel(*plan())(x, Wq, K_ext, V_ext, Wo)
```

```python
import dataclasses
import functools

import jax
import jax.numpy as jnp
from jax import lax
from jax.experimental import pallas as pl
from jax.experimental.pallas import tpu as pltpu

N_DEV = 4
B, SQ, DM, H, DH = 2, 256, 512, 4, 64
Q_SCALE = 0.125 * 1.4426950408889634
f32 = jnp.float32
bf16 = jnp.bfloat16
MESH = pl.DeviceIdType.MESH
ALL = frozenset(range(N_DEV))
GROUP_QB = {0: (0, 3), 1: (1, 2)}
NT = (((1,), (1,)), ((), ()))
PIECES = [(b, g, p) for b in range(2) for g in range(2) for p in range(2)]
PID = {pc: i for i, pc in enumerate(PIECES)}


def _add(xs):
    return functools.reduce(lambda u, v: u + v, xs)


def _allowed(qb, kb):
    return qb == kb or kb == 0 or (qb + kb) % 3 == 0


def _key_blocks(chip, g, u=None):
    qbs = GROUP_QB[g] if u is None else (GROUP_QB[g][u],)
    return [j for j in range(4) if any(_allowed(qb, 4 * chip + j) for qb in qbs)]


def _path(a, b, c, d, final):
    fs = frozenset
    return [(a, b, fs([a])), (d, c, fs([d])), (b, c, fs([a, b])), (c, b, fs([c, d])),
            (b, a, ALL if final else fs([b, c, d])), (c, d, ALL if final else fs([a, b, c]))]


SCHEME = {}
for _b in range(2):
    SCHEME[(_b, 0, 0)] = _path(3, 0, 1, 2, True)
    SCHEME[(_b, 0, 1)] = _path(2, 3, 0, 1, True)
    SCHEME[(_b, 1, 0)] = _path(0, 1, 2, 3, False)
    SCHEME[(_b, 1, 1)] = _path(1, 2, 3, 0, False)
MSGS = [(pc, s, d, ct) for pc in PIECES for (s, d, ct) in SCHEME[pc]]
Q_DST = {0: 1, 1: 3}


def _is_kv(m):
    return m[0][1] == 0 and len(m[3]) == 1


def _nblk(m):
    return len(_key_blocks(m[1], m[0][1]))


def _nsub(pc):
    return 8 if pc[1] == 1 else 2


def _parts(m):
    if _is_kv(m):
        return list(range(1 + _nblk(m)))
    if m[3] == ALL:
        return [0, 1]
    return ["s"] + list(range(_nsub(m[0])))


def _number(keys_by_chip):
    ids, cnt = {}, [0] * N_DEV
    for chip, key, size in keys_by_chip:
        ids[key] = cnt[chip]
        cnt[chip] += size
    return ids, max(cnt)


_SIZE = {m: 2 * (_nblk(m) if _is_kv(m) else 1) for m in MSGS if m[3] != ALL}
SSLOT, N_SSLOT = _number([(m[1], m, n) for m, n in _SIZE.items()])
RSLOT, N_RSLOT = _number([(m[2], m, n) for m, n in _SIZE.items()])
SSEM, N_SSEM = _number([(m[1], (m, u), 1) for m in MSGS for u in _parts(m)])
RSEM, N_RSEM = _number([(m[2], (m, u), 1) for m in MSGS for u in _parts(m)])


def _plan():
    both, lo, hi = (0, 1), (0, 1, 2, 3), (4, 5, 6, 7)
    loads, steps = {}, {}

    for c, f in ((1, 1), (3, 0)):
        s = 1 - f
        fp, sp = (f,), (s,)
        if c == 1:
            l0 = [("k", 0, fp, both), ("w", f), ("x", 0, 1), ("v", 0, fp, both),
                  ("k", 1, fp, both), ("x", 1, 1), ("v", 1, fp, both)]
            s0 = [("kprep", [(0, f, both)]), ("kvK", [(0, f)]), ("go",),
                  ("wq", fp), ("q", 0, 1, fp), ("s", 0, 1, fp, 2),
                  ("kprep", [(1, f, both)]), ("pv", 0, 1, fp, 2), ("flush", [(0, 1, f)]),
                  ("kvV", [(0, f)]), ("kvK", [(1, f)]), ("go",),
                  ("xc", 1, 1), ("roll", [(0, 1, f)]), ("q", 1, 1, fp), ("flush", [(0, 1, f)]),
                  ("kvV", [(1, f)]), ("s", 1, 1, fp, 2), ("go",)]
        else:
            l0 = [("vh", 0, f, 0), ("vh", 0, f, 1), ("k", 0, fp, both), ("w", f), ("x", 0, 1),
                  ("v", 1, fp, both), ("x", 1, 1), ("k", 1, fp, both)]
            s0 = [("kvV", [(0, f)], (0,)), ("go",), ("kvV", [(0, f)], (1,)), ("go",),
                  ("kprep", [(0, f, both)]), ("kvK", [(0, f)]), ("go",),
                  ("wq", fp), ("q", 0, 1, fp), ("kvV", [(1, f)]), ("go",), ("fence",),
                  ("s", 0, 1, fp, 2), ("pv", 0, 1, fp, 2), ("flush", [(0, 1, f)]),
                  ("xc", 1, 1), ("roll", [(0, 1, f)]), ("q", 1, 1, fp), ("flush", [(0, 1, f)]),
                  ("kprep", [(1, f, both)]), ("s", 1, 1, fp, 2), ("kvK", [(1, f)]), ("go",)]

        def relay(b, us, src=2):
            out = []
            for u in us:
                out += [("recv", [(b, 1, s, src, u)]), ("fwd", [(b, 1, s)])]
            return out

        loads[c] = l0 + [("k", 0, sp, both), ("v", 0, sp, both), ("k", 1, sp, both),
                         ("v", 1, sp, both), ("w", s), ("o",)]
        steps[c] = s0 + [
            ("kprep", [(0, s, both)]), ("pv", 1, 1, fp, 2), ("flush", [(1, 1, f)]),
            ("qrecv", 0), ("kvw", [(0, s, 0)]), ("roll", [(1, 1, f)]), ("s", 0, 0, sp), ("flush", [(1, 1, f)]),
            ("kvw", [(0, s, 1)]), ("kprep", [(1, s, both)]), ("pv", 0, 0, sp), ("flush", [(0, 0, s)]),
            ("wq", sp), ("q", 0, 1, sp),
            ("kvw", [(1, s, 0)]), ("qrecv", 1), ("s", 1, 0, sp), ("q", 1, 1, sp),
            ("kvw", [(1, s, 1)]), ("pv", 1, 0, sp), ("s", 0, 1, sp), ("s", 1, 1, sp), ("flush", [(1, 0, s)]),
            ("recv", [(0, 1, s, 0, "all")]), ("pv", 0, 1, sp), ("pv", 1, 1, sp), ("flush", [(0, 1, s)]),
            ("roll", [(0, 1, s), (1, 1, s)]), ("flush", [(0, 1, s)]),
            *relay(1, [lo], 0),
            *relay(0, [()] + [(u,) for u in range(6)]),
            *relay(1, [hi], 0),
            *relay(0, [(6,), (7,)]),
            *relay(1, [()] + [(u,) for u in range(8)]),
            ("recv", [(0, 0, s, 0, "all")]), ("wo",), ("flush", [(0, 0, s), (0, 1, s), (1, 1, s)]),
            ("recv", [(1, 0, s, 0, "all")]), ("flush", [(1, 0, s)]),
            ("out", 0, 1, sp), ("out", 1, 1, sp), ("out", 0, 0, sp), ("out", 1, 0, sp), ("drain", 6),
            ("recv", [(0, 0, f, 0, "all"), (0, 1, f, 2, "all")]),
            ("out", 0, 0, fp), ("flush", [(0, 1, f)]), ("out", 0, 1, fp),
            ("recv", [(1, 0, f, 0, "all"), (1, 1, f, 2, "all")]),
            ("out", 1, 0, fp), ("flush", [(1, 1, f)]), ("out", 1, 1, fp)]

    def pair(b, g):
        return [(b, g, 0), (b, g, 1)]

    def mid(b, g, us):
        return ("recv", [(b, g, 0, 1, us), (b, g, 1, 3, us)])

    loads[0] = [("w",), ("x", 0, 0), ("x", 1, 0), ("x", 0, 1), ("k", 0, both, both), ("v", 0, both, both),
                ("x", 1, 1), ("k", 1, both, both), ("v", 1, both, both), ("o",)]
    steps[0] = [
        ("wq", both), ("q", 0, 0, both), ("xc", 1, 0), ("q", 1, 0, both), ("qsend",),
        ("q", 0, 1, both), ("kprep", [(0, 0, both), (0, 1, both)]), ("s", 0, 1, both),
        ("pv", 0, 1, both), ("flush", pair(0, 1)),
        ("q", 1, 1, both), ("kprep", [(1, 0, both), (1, 1, both)]), ("s", 1, 1, both),
        ("pv", 1, 1, both), ("flush", pair(1, 1)),
        ("kvw", [(0, 1, 0), (0, 0, 0)]), ("s", 0, 0, both),
        ("kvw", [(0, 1, 1), (0, 0, 1), (1, 1, 0)]), ("wo", True), ("pv", 0, 0, both), ("s", 1, 0, (1,)),
        ("flush", [(0, 0, 1), (0, 0, 0)]),
        ("kvw", [(1, 1, 1)]), ("pv", 1, 0, (1,)), ("flush", [(1, 0, 1)]),
        ("kvw", [(1, 0, 0), (1, 0, 1)]), ("s", 1, 0, (0,), 2), ("pv", 1, 0, (0,)), ("flush", [(1, 0, 0)]),
        ("drain", 12),
        mid(0, 0, "all"), ("flush", pair(0, 0)), ("out", 0, 0, both),
        mid(1, 0, "all"), ("flush", pair(1, 0)), ("drain", 8),
        mid(0, 1, lo), ("out", 1, 0, (0,)), ("outp", 0, 1, 0),
        mid(0, 1, hi), ("out", 1, 0, (1,)), ("outp", 0, 1, 1),
        mid(1, 1, lo), ("outp", 1, 1, 0), ("drain", 0),
        mid(1, 1, hi), ("outp", 1, 1, 1)]

    def end(b, us):
        return ("recv", [(b, 1, 0, 3, us), (b, 1, 1, 1, us)])

    def fwd(b):
        return ("fwd", pair(b, 1))

    def kprep(b, t):
        return ("kprep", [(b, 0, (t,)), (b, 1, (t,))])

    loads[2] = [("k", 0, both, (0,)), ("v", 0, both, (0,)), ("k", 1, both, (0,)), ("v", 1, both, (0,)),
                ("w", 0), ("x", 0, 1), ("w", 1), ("k", 0, both, (1,)), ("v", 0, both, (1,)),
                ("xh", 1, 0), ("xh", 1, 1), ("k", 1, both, (1,)), ("v", 1, both, (1,)), ("o",)]
    steps[2] = [
        kprep(0, 0), ("kvK", [(0, 0), (0, 1)]), ("go",), ("kvV", [(0, 0), (0, 1)]), ("go",),
        kprep(1, 0), ("kvK", [(1, 0), (1, 1)]), ("go",), ("kvV", [(1, 0), (1, 1)]), ("go",),
        ("wq", (0,)), ("q", 0, 1, (0,)), ("wq", (1,)), ("q", 0, 1, (1,)),
        kprep(0, 1), ("s", 0, 1, both),
        ("need", ("xh", 1, 0)), end(0, (0, 1)), ("pv", 0, 1, both), ("qh", 1, 0), fwd(0), ("roll", pair(0, 1)),
        end(0, (2, 3, 4, 5)), fwd(0),
        kprep(1, 1), ("qh", 1, 1), ("s", 1, 1, both),
        end(0, (6, 7)), fwd(0),
        ("need", ("v", 1, 1, 1)), end(1, (0, 1)), ("pv", 1, 1, both), fwd(1), ("roll", pair(1, 1)),
        end(1, (2, 3, 4, 5)), fwd(1), end(1, (6, 7)), fwd(1),
        ("wo",),
        mid(0, 1, lo), fwd(0), mid(0, 1, hi), fwd(0), ("fence",), ("flush", pair(0, 1)),
        mid(1, 1, lo), fwd(1), ("fence",), ("out", 0, 1, both),
        mid(1, 1, hi), fwd(1), ("fence",), ("flush", pair(1, 1)), ("out", 1, 1, both), ("drain", 4),
        mid(0, 0, "all"), ("out", 0, 0, both),
        mid(1, 0, "all"), ("out", 1, 0, both)]
    return loads, steps


LOADS, STEPS = _plan()
N_LOAD_SEMS = 16


def _program(c, bar, x_hbm, wq_hbm, kt_hbm, vt_hbm, wo_hbm, out_ref,
             xb, wqb, ktb, vtb, wob, sbuf, sstat, rbuf, rstat, fin, qbuf,
             lsem, s_sem, r_sem, qs_sem, qr_sem, rdy):
    me = frozenset([c])

    loads, provides = [], {}

    def load(src, dst, *keys):
        cp = pltpu.make_async_copy(src, dst, lsem.at[len(loads)])
        cp.start()
        for k in keys:
            provides[k] = len(loads)
        loads.append(cp)

    for ck in LOADS[c]:
        kind = ck[0]
        if ck == ("w",):
            load(wq_hbm, wqb, ("w", 0), ("w", 1))
        elif kind == "w":
            cols = pl.ds(ck[1] * 128, 128)
            load(wq_hbm.at[:, cols], wqb.at[:, cols], ck)
        elif kind == "x" and ck[2] == 0:
            b = ck[1]
            load(x_hbm.at[pl.ds(b * 256, 64)], xb.at[b * 2, pl.ds(0, 64)])
            load(x_hbm.at[pl.ds(b * 256 + 192, 64)], xb.at[b * 2, pl.ds(64, 64)], ck)
        elif kind == "x":
            load(x_hbm.at[pl.ds(ck[1] * 256 + 64, 128)], xb.at[ck[1] * 2 + 1], ck)
        elif kind == "xh":
            _, b, u = ck
            load(x_hbm.at[pl.ds(b * 256 + 64 + u * 64, 64)], xb.at[b * 2 + 1, pl.ds(u * 64, 64)], ck)
        elif kind == "vh":
            _, b, p, h = ck
            rows = pl.ds(b * 256 + p * 128 + h * 64, 64)
            load(vt_hbm.at[rows], vtb.at[rows], ck, ("v", b, p, 0), ("v", b, p, 1))
        elif kind in ("k", "v"):
            _, b, ps, ts = ck
            src, dst = (kt_hbm, ktb) if kind == "k" else (vt_hbm, vtb)
            rows = pl.ds(b * 256 + ps[0] * 128, 128 * len(ps))
            keys = [(kind, b, p, t) for p in ps for t in ts]
            if len(ts) == 2:
                load(src.at[rows], dst.at[rows], *keys)
            else:
                cols = pl.ds(ts[0] * 128, 128)
                load(src.at[rows, cols], dst.at[rows, cols], *keys)
        else:
            load(wo_hbm, wob, ("o",))
    assert len(loads) <= N_LOAD_SEMS
    n_waited = [0]

    def need(*keys):
        last = max(provides[k] for k in keys)
        while n_waited[0] <= last:
            loads[n_waited[0]].wait()
            n_waited[0] += 1

    known = set()
    if c == 0:
        for d in (1, 3):
            pl.semaphore_signal(bar, inc=1, device_id=(d,), device_id_type=MESH)
    elif c == 2:
        pl.semaphore_wait(bar, 2)
        known.update((1, 3))
        for d in (1, 3):
            pl.semaphore_signal(rdy.at[2], inc=1, device_id=(d,), device_id_type=MESH)
    else:
        pl.semaphore_signal(bar, inc=1, device_id=(2,), device_id_type=MESH)
        pl.semaphore_wait(bar, 1)
        known.add(0)
        pl.semaphore_signal(rdy.at[c], inc=1, device_id=(0,), device_id_type=MESH)

    def know(d):
        if d not in known:
            pl.semaphore_wait(rdy.at[d], 1)
            known.add(d)

    lane64 = lax.broadcasted_iota(jnp.int32, (64, 128), 1) < 64
    lane128 = lax.broadcasted_iota(jnp.int32, (128, 128), 1) < 64
    lane1 = lane64[0:1]
    val = {}
    have = {pc + (u,): {} for pc in PIECES for u in range(_nsub(pc))}
    lses = {pc: {} for pc in PIECES}
    final, sent, got, done = set(), set(), set(), set()
    queue, started = [], []

    def views(m, u):
        pc, _, _, ct = m
        if ct == ALL:
            r = fin.at[PID[pc], pl.ds(u * 64, 64)]
            return r, r
        if u == "s":
            return sstat.at[SSLOT[m] // 2], rstat.at[RSLOT[m] // 2]
        if _is_kv(m):
            off, n = (0, _nblk(m) * 64) if u == 0 else ((_nblk(m) + u - 1) * 64, 64)
        else:
            n = 128 // _nsub(pc)
            off = u * n
        return sbuf.at[pl.ds(SSLOT[m] * 64 + off, n)], rbuf.at[pl.ds(RSLOT[m] * 64 + off, n)]

    def rdma(src, dst, ssem, rsem, peer):
        return pltpu.make_async_remote_copy(src, dst, ssem, rsem, device_id=(peer,), device_id_type=MESH)

    def enqueue(m, u):
        sent.add((m, u))
        queue.append((m, u))

    def go():
        for m, _ in queue:
            know(m[2])
        for m, u in queue:
            src, dst = views(m, u)
            cp = rdma(src, dst, s_sem.at[SSEM[(m, u)]], r_sem.at[RSEM[(m, u)]], m[2])
            cp.start()
            started.append(cp)
        queue.clear()

    def wait_msgs(lst):
        for m, u in lst:
            if (m, u) not in got:
                dst = views(m, u)[1]
                rdma(dst, dst, s_sem.at[0], r_sem.at[RSEM[(m, u)]], m[1]).wait_recv()
                got.add((m, u))

    def kv_in(pc):
        return [m for m in MSGS if m[0] == pc and m[2] == c and _is_kv(m)]

    def put(pc, h, ct, o):
        k = _nsub(pc) // 2
        for i in range(k):
            have[pc + (k * h + i,)][ct] = o[(64 // k) * i:(64 // k) * (i + 1)]

    def cover(held, ct):
        rem, parts = set(ct), []
        for k in sorted(held, key=lambda k: -len(k)):
            if k <= rem:
                parts.append(k)
                rem -= k
        return None if rem else parts

    def weights(pc, ct):
        key = ("wts", pc, ct)
        if key not in val:
            parts = cover(lses[pc], ct)
            if parts is None:
                return None
            if len(parts) == 1:
                val[key] = (parts, None)
            else:
                ls = [lses[pc][k] for k in parts]
                m = functools.reduce(jnp.maximum, ls)
                a = [jnp.exp2(v - m) for v in ls]
                s = _add(a)
                inv = 1.0 / s
                val[key] = (parts, [ai * inv for ai in a])
                if ct != ALL:
                    lses[pc][ct] = m + jnp.log2(s)
        return val[key]

    def merged(pc, u, ct):
        hv = have[pc + (u,)]
        if ct in hv:
            return hv[ct]
        pw = weights(pc, ct)
        if pw is None or len(pw[0]) == 1:
            return None
        vals = [merged(pc, u, k) for k in pw[0]]
        if any(v is None for v in vals):
            return None
        h = u * 2 // _nsub(pc)
        hv[ct] = _add([w[:, h * 128:(h + 1) * 128] * v for w, v in zip(pw[1], vals)])
        return hv[ct]

    def stage(pc, finalise):
        outs = [m for m in MSGS if m[0] == pc and m[1] == c and not _is_kv(m)]
        for m in outs:
            if m[3] != ALL and (m, "s") not in sent and weights(pc, m[3]) is not None:
                sstat[SSLOT[m] // 2] = lses[pc][m[3]]
                enqueue(m, "s")
        n = 128 // _nsub(pc)
        for u in range(_nsub(pc)):
            for m in outs:
                if m[3] != ALL and (m, u) not in sent:
                    o = merged(pc, u, m[3])
                    if o is not None:
                        sbuf[pl.ds(SSLOT[m] * 64 + u * n, n)] = o.astype(bf16)
                        enqueue(m, u)
        if (finalise and pc not in final
                and all(cover(have[pc + (u,)], ALL) is not None for u in range(_nsub(pc)))):
            o = [merged(pc, u, ALL) for u in range(_nsub(pc))]
            fin[PID[pc]] = jnp.concatenate(o, axis=0).T.astype(bf16)
            final.add(pc)
            for m in outs:
                if m[3] == ALL:
                    enqueue(m, 0)
                    enqueue(m, 1)

    def softmax(s):
        m = jnp.max(s, axis=0, keepdims=True)
        pt = jnp.exp2(s - m)
        l = jnp.sum(pt, axis=0, keepdims=True)
        return pt, 1.0 / l, m + jnp.log2(l)

    def scores(k, q):
        return lax.dot_general(k, q, NT, preferred_element_type=f32)

    def matmul(a, b_):
        return jnp.dot(a, b_, preferred_element_type=f32)

    def head_tiles(qp):
        return jnp.concatenate([jnp.where(lane128, qp, 0.0), jnp.where(lane128, 0.0, qp)], axis=0).astype(bf16)

    def block_tile(qp, u):
        q0, q1 = jnp.where(lane64, qp, 0.0), jnp.where(lane64, 0.0, qp)
        return jnp.concatenate([q0, q1] if u == 0 else [q1, q0], axis=0).astype(bf16)

    def accumulate(b, g, terms):
        if ("acc", b, g) in val:
            terms = terms + [val.pop(("acc", b, g))]
        o, n = _add([t for t, _ in terms]), sum(k for _, k in terms)
        if n < H:
            val[("acc", b, g)] = (o, n)
        else:
            if g == 0:
                out_ref[b, 0:64, :] = o[0:64]
                out_ref[b, 192:256, :] = o[64:128]
            else:
                out_ref[b, 64:192, :] = o
            done.add((b, g))

    zero = jnp.zeros((64, 128), f32)

    for step in STEPS[c]:
        op = step[0]
        by_block = op in ("q", "s", "pv") and step[2] == 1 and c != 0
        if op == "need":
            need(*step[1:])
        elif op == "kprep":
            need(*[("k", b, p, t) for b, p, ts in step[1] for t in ts])
            for b, p, ts in step[1]:
                kk = ktb[pl.ds(b * 256 + p * 128, 128), pl.ds(ts[0] * 128, 128 * len(ts))].T
                for i in range(2 * len(ts)):
                    val[("k", b, p, 2 * ts[0] + i)] = kk[i * 64:(i + 1) * 64]
        elif op == "kvK":
            for b, p in step[1]:
                m, = [m for m in MSGS if m[0] == (b, 0, p) and m[1] == c]
                for i, j in enumerate(_key_blocks(c, 0)):
                    sbuf[pl.ds((SSLOT[m] + i) * 64, 64)] = val[("k", b, p, j)].astype(bf16)
                enqueue(m, 0)
        elif op == "kvV":
            js = _key_blocks(c, 0)
            heads = step[2] if len(step) > 2 else (0, 1)
            if len(step) > 2:
                need(*[("vh", b, p, h) for b, p in step[1] for h in heads])
            else:
                need(*[("v", b, p, j // 2) for b, p in step[1] for j in js])
            for b, p in step[1]:
                m, = [m for m in MSGS if m[0] == (b, 0, p) and m[1] == c]
                if len(js) == 1:
                    v = vtb[pl.ds(b * 256 + p * 128, 128), pl.ds((js[0] // 2) * 128, 128)]
                    v0, v1 = v[0:64], v[64:128]
                    if js[0] % 2 == 1:
                        v0 = pltpu.roll(v0, 64, 1)
                    else:
                        v1 = pltpu.roll(v1, 64, 1)
                    sbuf[pl.ds((SSLOT[m] + 1) * 64, 64)] = jnp.where(lane64, v0, v1).astype(bf16)
                    enqueue(m, 1)
                else:
                    assert js == [0, 3]
                    for h in heads:
                        rows = pl.ds(b * 256 + p * 128 + h * 64, 64)
                        sbuf[pl.ds((SSLOT[m] + 2 + h) * 64, 64)] = jnp.where(
                            lane64, vtb[rows, 0:128], vtb[rows, 128:256]).astype(bf16)
                        enqueue(m, 1 + h)
        elif op == "kvw":
            wait_msgs([(m, u) for b, p, part in step[1] for m in kv_in((b, 0, p))
                       for u in (_parts(m)[:1] if part == 0 else _parts(m)[1:])])
        elif op == "wq":
            need(*[("w", p) for p in step[1]])
            for p in step[1]:
                val[("w", p)] = wqb[:, pl.ds(p * 128, 128)].astype(bf16)
        elif op in ("xc", "q"):
            b, g = step[1:3]
            if ("x", b, g) not in val:
                need(("x", b, g))
                val[("x", b, g)] = xb[b * 2 + g].astype(bf16)
            for p in (step[3] if op == "q" else ()):
                qp = matmul(val[("x", b, g)], val[("w", p)]) * Q_SCALE
                val[("qraw", b, g, p)] = qp
                if by_block:
                    for u in range(2):
                        val[("q", b, g, p, u)] = block_tile(qp[u * 64:(u + 1) * 64], u)
                else:
                    val[("q", b, g, p)] = head_tiles(qp)
        elif op == "qh":
            _, b, u = step
            need(("xh", b, u))
            xv = xb[b * 2 + 1, pl.ds(u * 64, 64)].astype(bf16)
            for p in range(2):
                val[("q", b, 1, p, u)] = block_tile(matmul(xv, val[("w", p)]) * Q_SCALE, u)
        elif op == "qsend":
            for i in range(4):
                qbuf[i] = val[("qraw", i // 2, 0, i % 2)].astype(bf16)
            for d in Q_DST.values():
                know(d)
            for i in range(4):
                cp = rdma(qbuf.at[i], qbuf.at[i], qs_sem.at[i], qr_sem.at[i], Q_DST[i % 2])
                cp.start()
                started.append(cp)
        elif op == "qrecv":
            p, = [p for p, d in Q_DST.items() if d == c]
            i = step[1] * 2 + p
            rdma(qbuf.at[i], qbuf.at[i], qs_sem.at[i], qr_sem.at[i], 0).wait_recv()
            val[("q", step[1], 0, p)] = head_tiles(qbuf[i].astype(f32))
        elif op == "s" and by_block:
            _, b, g, ps = step[:4]
            raw = {}
            for p in ps:
                for u in range(2):
                    ks = [val[("k", b, p, j)] for j in _key_blocks(c, g, u)]
                    q = val[("q", b, g, p, u)]
                    if len(step) > 4:
                        raw[(p, u)] = jnp.concatenate([scores(k.astype(bf16), q) for k in ks], axis=0)
                    else:
                        raw[(p, u)] = scores(jnp.concatenate(ks, axis=0).astype(bf16), q)
            for p in ps:
                val[("p", b, g, p)] = [softmax(raw[(p, u)]) for u in range(2)]
        elif op == "pv" and by_block:
            _, b, g, ps = step[:4]
            need(*[("v", b, p, t) for p in ps for t in range(2)])
            for p in ps:
                res = val[("p", b, g, p)]
                rows = pl.ds(b * 256 + p * 128, 128)
                oo = []
                for u in range(2):
                    js = _key_blocks(c, g, u)
                    pt = res[u][0]
                    if len(js) == 2:
                        assert js == [0, 3]
                        vv = jnp.where(lane128, vtb[rows, 0:128], vtb[rows, 128:256])
                    else:
                        vv = vtb[rows, pl.ds((js[0] // 2) * 128, 128)]
                        pt = jnp.concatenate([pt, zero] if js[0] % 2 == 0 else [zero, pt], axis=0)
                    ptb = pt.astype(bf16)
                    if len(step) > 4:
                        oo.append([matmul(vv[h * 64:(h + 1) * 64].astype(bf16), ptb) for h in range(2)])
                    else:
                        o = matmul(vv.astype(bf16), ptb)
                        oo.append([o[0:64], o[64:128]])
                lses[(b, g, p)][me] = jnp.concatenate(
                    [jnp.where(lane1, res[0][2], res[1][2]),
                     pltpu.roll(jnp.where(lane1, res[1][2], res[0][2]), 64, 1)], axis=1)
                put((b, g, p), 0, me,
                    jnp.where(lane64, oo[0][0], oo[1][0]) * jnp.where(lane1, res[0][1], res[1][1]))
                val[("swapped", b, g, p)] = (jnp.where(lane64, oo[1][1], oo[0][1])
                                             * jnp.where(lane1, res[1][1], res[0][1]))
        elif op == "roll":
            for pc in step[1]:
                put(pc, 1, me, pltpu.roll(val.pop(("swapped",) + pc), 64, 1))
        elif op == "s":
            _, b, g, ps = step[:4]
            split = step[4] if len(step) > 4 else 1
            js = _key_blocks(c, g)
            assert js == _key_blocks(c, g, 0) == _key_blocks(c, g, 1)
            wait_msgs([(m, 0) for p in ps for m in kv_in((b, g, p))])
            raw = {}
            for p in ps:
                q = val[("q", b, g, p)]
                kall = jnp.concatenate([val[("k", b, p, j)] for j in js], axis=0)
                n = kall.shape[0] // split
                raw[p] = [scores(kall[i * n:(i + 1) * n].astype(bf16), q) for i in range(split)]
                raw[p] += [scores(rbuf[pl.ds(RSLOT[m] * 64, _nblk(m) * 64)], q) for m in kv_in((b, g, p))]
            for p in ps:
                val[("p", b, g, p)] = softmax(jnp.concatenate(raw[p], axis=0))
        elif op == "pv":
            _, b, g, ps = step[:4]
            js = _key_blocks(c, g)
            need(*[("v", b, p, j // 2) for p in ps for j in js])
            wait_msgs([(m, u) for p in ps for m in kv_in((b, g, p)) for u in _parts(m)[1:]])
            for p in ps:
                pc = (b, g, p)
                pt, inv, lse = val[("p", b, g, p)]
                ct = frozenset([c] + [m[1] for m in kv_in(pc)])
                for h in range(2):
                    vrows = pl.ds(b * 256 + p * 128 + h * 64, 64)
                    cols = slice(h * 128, (h + 1) * 128)
                    blk = {j: pt[i * 64:(i + 1) * 64, cols] for i, j in enumerate(js)}
                    terms = []
                    if js == [0, 3]:
                        terms.append((jnp.where(lane64, vtb[vrows, 0:128], vtb[vrows, 128:256]).astype(bf16),
                                      jnp.concatenate([blk[0], blk[3]], axis=0)))
                    else:
                        for t in sorted({j // 2 for j in js}):
                            terms.append((vtb[vrows, pl.ds(t * 128, 128)].astype(bf16),
                                          jnp.concatenate([blk.get(2 * t, zero), blk.get(2 * t + 1, zero)], axis=0)))
                    off = len(js) * 64
                    for m in kv_in(pc):
                        pr = pt[off:off + _nblk(m) * 64, cols]
                        off += _nblk(m) * 64
                        if _nblk(m) == 1:
                            terms.append((rbuf[pl.ds((RSLOT[m] + 1) * 64, 64)],
                                          jnp.concatenate([pr, zero] if h == 0 else [zero, pr], axis=0)))
                        else:
                            terms.append((rbuf[pl.ds((RSLOT[m] + 2 + h) * 64, 64)], pr))
                    put(pc, h, ct, _add([matmul(vv, pp.astype(bf16)) for vv, pp in terms]) * inv[:, cols])
                lses[pc][ct] = lse
        elif op == "recv":
            lst = []
            for b, g, p, src, us in step[1]:
                m, = [m for m in MSGS if m[:3] == ((b, g, p), src, c)]
                us = [u for u in _parts(m) if u == "s" or us == "all" or u in us]
                lst += [(m, u) for u in us if (m, u) not in got]
            wait_msgs(lst)
            for m, u in lst:
                if m[3] == ALL:
                    final.add(m[0])
                elif u == "s":
                    lses[m[0]][m[3]] = rstat[RSLOT[m] // 2]
                else:
                    n = 128 // _nsub(m[0])
                    have[m[0] + (u,)][m[3]] = rbuf[pl.ds(RSLOT[m] * 64 + u * n, n)].astype(f32)
        elif op in ("flush", "fwd"):
            for pc in step[1]:
                stage(pc, op == "flush")
            go()
        elif op == "go":
            go()
        elif op == "fence":
            pl.semaphore_signal(rdy.at[c], inc=1)
            pl.semaphore_wait(rdy.at[c], 1)
        elif op == "drain":
            n = len(started) - step[1]
            for cp in started[:n]:
                cp.wait_send()
            del started[:n]
        elif op == "wo":
            need(("o",))
            val["wo"] = [wob[0:128, :].astype(bf16), wob[128:256, :].astype(bf16)]
            if len(step) > 1:
                val["wop"] = [jnp.concatenate([wob[h * 64:(h + 1) * 64, :], wob[128 + h * 64:192 + h * 64, :]],
                                              axis=0).astype(bf16) for h in range(2)]
        elif op == "out":
            _, b, g, ps = step
            assert all((b, g, p) in final for p in ps)
            accumulate(b, g, [(matmul(fin[PID[(b, g, p)]], val["wo"][p]), 2) for p in ps])
        elif op == "outp":
            _, b, g, h = step
            k = _nsub((b, g, 0)) // 2
            o = [merged((b, g, p), u, ALL) for p in range(2) for u in range(h * k, (h + 1) * k)]
            accumulate(b, g, [(matmul(jnp.concatenate(o, axis=0).T.astype(bf16), val["wop"][h]), 2)])
        else:
            raise ValueError(step)

    for cp in started:
        cp.wait_send()

    assert not queue and n_waited[0] == len(loads) and len(done) == 4
    assert known == {(c + 1) % N_DEV, (c + 3) % N_DEV}
    assert sent == {(m, u) for m in MSGS if m[1] == c for u in _parts(m)}
    assert got == {(m, u) for m in MSGS if m[2] == c for u in _parts(m)}


def _compiler_params():
    want = dict(collective_id=0, disable_bounds_checks=True, disable_semaphore_checks=True)
    names = {f.name for f in dataclasses.fields(pltpu.CompilerParams)}
    return pltpu.CompilerParams(**{k: v for k, v in want.items() if k in names})


def pallas_dist_sparse_attn_blocksparse_kvseq_b2_sq256_skv256_hq4_dh64_kernel(
    x: jax.Array,
    Wq: jax.Array,
    K_ext: jax.Array,
    V_ext: jax.Array,
    Wo: jax.Array,
):
    kt = jnp.transpose(K_ext, (0, 2, 3, 1)).reshape(B * H * DH, SQ)
    vt = jnp.transpose(V_ext, (0, 2, 3, 1)).reshape(B * H * DH, SQ)
    x2 = x.reshape(B * SQ, DM)

    def body(*refs):
        my = lax.axis_index("i")
        bar = pltpu.get_barrier_semaphore()
        for c in (2, 3, 1, 0):
            pl.when(my == c)(functools.partial(_program, c, bar, *refs))

    return pl.pallas_call(
        body,
        out_shape=jax.ShapeDtypeStruct((B, SQ, DM), f32),
        in_specs=[pl.BlockSpec(memory_space=pl.ANY)] * 5,
        out_specs=pl.BlockSpec(memory_space=pltpu.VMEM),
        scratch_shapes=[
            pltpu.VMEM((4, 128, DM), f32),
            pltpu.VMEM((DM, H * DH), f32),
            pltpu.VMEM((B * H * DH, SQ), f32),
            pltpu.VMEM((B * H * DH, SQ), f32),
            pltpu.VMEM((H * DH, DM), f32),
            pltpu.VMEM((N_SSLOT * 64, 128), bf16),
            pltpu.VMEM((N_SSLOT // 2, 1, 256), f32),
            pltpu.VMEM((N_RSLOT * 64, 128), bf16),
            pltpu.VMEM((N_RSLOT // 2, 1, 256), f32),
            pltpu.VMEM((8, 128, 128), bf16),
            pltpu.VMEM((4, 128, 128), bf16),
            pltpu.SemaphoreType.DMA((N_LOAD_SEMS,)),
            pltpu.SemaphoreType.DMA((N_SSEM,)),
            pltpu.SemaphoreType.DMA((N_RSEM,)),
            pltpu.SemaphoreType.DMA((4,)),
            pltpu.SemaphoreType.DMA((4,)),
            pltpu.SemaphoreType.REGULAR((N_DEV,)),
        ],
        compiler_params=_compiler_params(),
    )(x2, Wq, kt, vt, Wo)
```
